```python
import numpy as np

kernel_name = "dist_pipemlp_pp2tp2_xy_b4096_d256_h512"

def setup_inputs():
    x_padded = np.zeros((2, 4096, 256), dtype=np.float32)
    x_padded[0] = np.random.randn(4096, 256).astype(np.float32)
    Win = np.random.randn(4, 256, 1024).astype(np.float32)
    Wout = np.random.randn(4, 1024, 256).astype(np.float32)
    return {"x_padded": x_padded, "Win": Win, "Wout": Wout}

def reference(x_padded, Win, Wout):
    a = x_padded[0]
    for k in range(4):
        h = a @ Win[k]
        h = np.maximum(h, 0.0)
        a = h @ Wout[k]
    out = np.zeros_like(x_padded)
    out[1] = a
    return out
```

```python
import contextlib
import jax
import jax.numpy as jnp
from jax import lax
from jax.experimental import pallas as pl
from jax.experimental.pallas import tpu as pltpu

BF = jnp.bfloat16
F32 = jnp.float32
MESH = pl.DeviceIdType.MESH

NB = 4096
DM = 256
HH = 512
HALF = 2048
CH = 64
NCH = HALF // CH


def _mlp(a, win, wout):
    h = jnp.dot(a, win, preferred_element_type=F32)
    h = jnp.maximum(h, 0.0).astype(BF)
    return jnp.dot(h, wout, preferred_element_type=F32)


def _split(total, sizes, base=0):
    out, s, i = [], 0, 0
    while s < total:
        z = min(sizes[min(i, len(sizes) - 1)], total - s)
        out.append((base + s, z))
        s += z
        i += 1
    return out


DEFAULT = dict(
    fill=192,
    n1=6,
    p2=(128, 448),
    g0=8,
    rel1=(6, 7),
    rel2=(10,),
    kf=14,
    relp=64,
    last_split=(64, 32, 32),
    conv_at={8: 1, 10: 2, 12: 3, 13: 4, 14: 5, 15: 6},
    scopes=False,
)


def make(**kw):
    cfg = dict(DEFAULT)
    cfg.update(kw)
    FILL = cfg["fill"]
    N1 = cfg["n1"]
    G0 = cfg["g0"]
    KF = cfg["kf"]
    P1R = N1 * 128
    assert FILL + sum(cfg["p2"]) == P1R
    REL1 = list(cfg["rel1"])
    REL2 = list(cfg["rel2"])
    RELB = REL1 + REL2
    Z = 128 * len(RELB)
    RELP = []
    for bi, b in enumerate(RELB):
        sizes = (cfg["relp"],)
        if bi == len(RELB) - 1:
            sizes = cfg.get("rel_last", (64, 32, 32))
        for (a, n) in _split(128, sizes):
            RELP.append((bi * 128 + a, n, b * 128 + a))
    NREL = len(RELP)
    NREL1 = sum(1 for p in RELP if p[0] < 128 * len(REL1))
    DIR = _split(P1R - FILL, cfg["p2"], FILL)
    ND2 = len(DIR)
    blk_msgs = {}
    for b in range(N1, 16):
        if b in RELB:
            continue
        parts = _split(128, cfg["last_split"], b * 128) if b == 15 else [(b * 128, 128)]
        blk_msgs[b] = list(range(len(DIR), len(DIR) + len(parts)))
        DIR += parts
    NDIR = len(DIR)
    NDROWS = sum(n for _, n in DIR)

    WINP = _split(DM, cfg.get("win_pieces", (32, 96, 128)))

    def scope(name):
        if cfg["scopes"]:
            return jax.named_scope(name)
        return contextlib.nullcontext()

    def body(x_hbm, win_hbm, wout_hbm, out,
             big, pown, zbuf, wfin, wfout, wbin, wbout,
             ysend, yrecv, xsend, xrecv):
        def scoped(ld, wr, yr, xr, ss):
            inner(x_hbm, win_hbm, wout_hbm, out, big, pown, zbuf, wfin, wfout, wbin, wbout,
                  ysend, yrecv, xsend, xrecv, ld, wr, yr, xr, ss)
        pl.run_scoped(
            scoped,
            pltpu.SemaphoreType.DMA((32,)),
            pltpu.SemaphoreType.DMA((8,)),
            pltpu.SemaphoreType.DMA((max(NCH + NREL, NDIR + 1),)),
            pltpu.SemaphoreType.DMA((NCH + NREL,)),
            pltpu.SemaphoreType.DMA((16,)),
        )

    def inner(x_hbm, win_hbm, wout_hbm, out,
              big, pown, zbuf, wfin, wfout, wbin, wbout,
              ysend, yrecv, xsend, xrecv,
              ld, wr, yr, xr, ss):
        mx = lax.axis_index("x")
        my = lax.axis_index("y")
        ynb = (mx, 1 - my)
        xnb = (1 - mx, my)
        own0 = my * HALF
        oth0 = (1 - my) * HALF
        bar = pltpu.get_barrier_semaphore()

        def rcopy(src, dst, ssem, rsem, dev):
            return pltpu.make_async_remote_copy(
                src_ref=src, dst_ref=dst, send_sem=ssem, recv_sem=rsem,
                device_id=dev, device_id_type=MESH)

        hb = [1 - mx, mx]
        NP = len(WINP)
        L_WO0, L_WI1, L_WO1, L_X = NP, NP + 1, NP + 2, NP + 3

        def ld_win(slot, r0, n, k):
            return pltpu.make_async_copy(
                win_hbm.at[hb[slot], pl.ds(r0, n), :], wfin.at[slot, pl.ds(r0, n), :], ld.at[k])

        def ld_wout(slot, k):
            return pltpu.make_async_copy(wout_hbm.at[hb[slot]], wfout.at[slot], ld.at[k])

        def cv_win(slot, r0, n):
            wbin[slot, pl.ds(r0, n), pl.ds(0, HH)] = wfin[slot, pl.ds(r0, n), :].astype(BF)

        def cv_wout(slot):
            wbout[slot, pl.ds(0, HH), :] = wfout[slot].astype(BF)

        def y_win(slot, r0=0, n=DM):
            return rcopy(wbin.at[slot, pl.ds(r0, n), pl.ds(0, HH)],
                         wbin.at[slot, pl.ds(r0, n), pl.ds(HH, HH)],
                         ss.at[2 * slot], wr.at[2 * slot], ynb)

        def y_wout(slot):
            return rcopy(wbout.at[slot, pl.ds(0, HH), :], wbout.at[slot, pl.ds(HH, HH), :],
                         ss.at[2 * slot + 1], wr.at[2 * slot + 1], ynb)

        def x_win(half, r0=0, n=DM):
            return rcopy(wbin.at[0, pl.ds(r0, n), pl.ds(half * HH, HH)],
                         wbin.at[2, pl.ds(r0, n), pl.ds(half * HH, HH)],
                         ss.at[4 + 2 * half], wr.at[4 + 2 * half], xnb)

        def x_wout(half):
            return rcopy(wbout.at[0, pl.ds(half * HH, HH), :], wbout.at[2, pl.ds(half * HH, HH), :],
                         ss.at[5 + 2 * half], wr.at[5 + 2 * half], xnb)

        S_Y, S_X, S_RY, S_RX, S_F, S_Z = 8, 9, 10, 11, 12, 13
        RB = 1024

        def xload(i):
            base = oth0 if i % 2 == 0 else own0
            off = pl.multiple_of(base + (i // 2) * 256, 256)
            return pltpu.make_async_copy(
                x_hbm.at[0, pl.ds(off, 256), :], big.at[pl.ds(i * 256, 256), :], ld.at[L_X + i // 2])

        with scope("s0_pro"):
            pl.semaphore_signal(bar, inc=1, device_id=ynb, device_id_type=MESH)
            ld_win(0, *WINP[0], 0).start()
            ld_win(0, *WINP[1], 1).start()

            @pl.when(mx == 0)
            def _():
                pl.semaphore_signal(bar, inc=1, device_id=xnb, device_id_type=MESH)
                ld_win(1, 0, DM, L_WI1).start()
                xload(0).start()
                xload(1).start()
                ld_wout(1, L_WO1).start()
                for j in range(2, NP):
                    ld_win(0, *WINP[j], j).start()
                xload(2).start()
                xload(3).start()
                ld_wout(0, L_WO0).start()
                for i in range(4, 16):
                    xload(i).start()

            @pl.when(mx == 1)
            def _():
                for j in range(2, NP):
                    ld_win(0, *WINP[j], j).start()
                ld_wout(0, L_WO0).start()
                ld_win(1, 0, DM, L_WI1).start()
                ld_wout(1, L_WO1).start()

            ld_win(0, *WINP[0], 0).wait()
            cv_win(0, *WINP[0])
            pl.semaphore_wait(bar, 1 + mx)
            y_win(0, *WINP[0]).start()
            ld_win(0, *WINP[1], 1).wait()
            cv_win(0, *WINP[1])
            y_win(0, *WINP[1]).start()

        @pl.when(mx == 0)
        def _stage0():
            with scope("s0_init"):
                ld_win(1, 0, DM, L_WI1).wait()
                cv_win(1, 0, DM)
                ld_wout(1, L_WO1).wait()
                cv_wout(1)

            def xwait(i):
                r = i * 512 if isinstance(i, int) else pl.multiple_of(i * 512, 512)
                pltpu.make_async_copy(
                    big.at[pl.ds(r, 512), :], big.at[pl.ds(r, 512), :], ld.at[L_X + i]).wait()

            def l0(row, n):
                a = big[pl.ds(row, n), :].astype(BF)
                return _mlp(a, wbin[1, :, pl.ds(0, HH)], wbout[1, pl.ds(0, HH), :])

            def psend(k):
                r = k * CH if isinstance(k, int) else pl.multiple_of(k * CH, CH)
                return rcopy(ysend.at[pl.ds(r, CH), :], yrecv.at[pl.ds(r, CH), :],
                             ss.at[S_Y], yr.at[k], ynb)

            def l0_blk(i):
                dyn = not isinstance(i, int)
                r = pl.multiple_of(i * 512, 512) if dyn else i * 512
                q = pl.multiple_of(i * 256, 256) if dyn else i * 256
                p = l0(r, 512)
                ysend[pl.ds(q, 256), :] = p[:256].astype(BF)
                pown[pl.ds(q, 256), :] = p[256:]

            with scope("s0_l0"):
                xwait(0)
                for j in range(2, NP):
                    ld_win(0, *WINP[j], j).wait()
                for j in range(2, NP):
                    cv_win(0, *WINP[j])
                    y_win(0, *WINP[j]).start()
                l0_blk(0)
                ld_wout(0, L_WO0).wait()
                xwait(1)
                cv_wout(0)
                y_wout(0).start()
                for k in range(4):
                    psend(k).start()

                def it(i, c):
                    l0_blk(i)
                    xwait(i + 1)
                    for q in range(4):
                        psend(i * 4 + q).start()
                    return c
                lax.fori_loop(1, 7, it, 0)
                zbuf[...] = jnp.zeros_like(zbuf)
                for i in range(NB // 512):
                    pltpu.make_async_copy(zbuf, out.at[0, pl.ds(i * 512, 512), :], ss.at[S_Z]).start()

            with scope("s0_wait_w1"):
                y_win(0).wait_recv()
                y_wout(0).wait_recv()
                x_win(0).wait_recv()

            def chunk(k, g3):
                r = pl.multiple_of(k * CH, CH)
                psend(k).wait_recv()
                a = (pown[pl.ds(r, CH), :] + yrecv[pl.ds(r, CH), :].astype(F32)).astype(BF)
                a = _mlp(a, wbin[0], wbout[0]).astype(BF)
                if g3:
                    a = _mlp(a, wbin[2], wbout[2]).astype(BF)
                xsend[pl.ds(r, CH), :] = a
                rcopy(xsend.at[pl.ds(r, CH), :], xrecv.at[pl.ds(r, CH), :],
                      ss.at[S_X], xr.at[k], xnb).start()

            def pair_late_oth(j, c):
                chunk(2 * j, False)
                r = pl.multiple_of(j * CH, CH)
                ysend[pl.ds(7 * 256 + r, CH), :] = l0(7 * 512 + r, CH).astype(BF)
                psend(28 + j).start()
                chunk(2 * j + 1, False)
                return c

            def pair_late_own(j, c):
                chunk(2 * j, False)
                r = pl.multiple_of((j - 4) * CH, CH)
                pown[pl.ds(7 * 256 + r, CH), :] = l0(7 * 512 + 256 + r, CH)
                chunk(2 * j + 1, False)
                return c

            def pair_plain(j, c):
                chunk(2 * j, False)
                chunk(2 * j + 1, False)
                return c

            def pair_g3(j, c):
                chunk(2 * j, False)
                chunk(2 * j + 1, True)
                return c

            def rel_in(lo, hi, sem):
                return rcopy(ysend.at[pl.ds(lo, hi - lo), :], xrecv.at[pl.ds(lo, hi - lo), :],
                             ss.at[S_RX], xr.at[sem], xnb)

            def rel_y(j):
                a, n, _ = RELP[j]
                return rcopy(xrecv.at[pl.ds(a, n), :], xrecv.at[pl.ds(RB + a, n), :],
                             ss.at[S_RY], yr.at[NCH + j], ynb)

            def rel_x(j):
                a, n, o = RELP[j]
                return rcopy(xrecv.at[pl.ds(RB + a, n), :], yrecv.at[pl.ds(o, n), :],
                             ss.at[S_RX], xr.at[NCH + j], xnb)

            with scope("s0_p2a"):
                lax.fori_loop(0, 4, pair_late_oth, 0)
                lax.fori_loop(4, 8, pair_late_own, 0)
                if G0 > 8:
                    lax.fori_loop(8, G0, pair_plain, 0)
            with scope("s0_wait_w2"):
                x_wout(0).wait_recv()
                x_win(1).wait_recv()
                x_wout(1).wait_recv()
            with scope("s0_p2b"):
                lax.fori_loop(G0, KF, pair_g3, 0)
            with scope("s0_relay1"):
                if REL1:
                    rel_in(0, 128 * len(REL1), 0).wait_recv()
                    for j in range(NREL1):
                        rel_y(j).start()
            with scope("s0_p2c"):
                lax.fori_loop(KF, 16, pair_g3, 0)
            with scope("s0_relay2"):
                if REL2:
                    rel_in(128 * len(REL1), Z, 1).wait_recv()
                    for j in range(NREL1, NREL):
                        rel_y(j).start()
                for j in range(NREL):
                    rel_y(j).wait_recv()
                    rel_x(j).start()

        @pl.when(mx == 1)
        def _stage1():
            a3 = xsend
            with scope("s1_init"):
                x_win(0, 0, WINP[2][0]).start()
                for j in range(2, NP):
                    ld_win(0, *WINP[j], j).wait()
                    cv_win(0, *WINP[j])
                    y_win(0, *WINP[j]).start()
                    x_win(0, *WINP[j]).start()
                ld_wout(0, L_WO0).wait()
                cv_wout(0)
                y_wout(0).start()
                x_wout(0).start()
                ld_win(1, 0, DM, L_WI1).wait()
                cv_win(1, 0, DM)
                y_win(1).start()
                ld_wout(1, L_WO1).wait()
                cv_wout(1)
                y_wout(1).start()
            with scope("s1_wait_w2"):
                y_win(0).wait_recv()
                x_win(1).start()
                y_wout(0).wait_recv()
                x_wout(1).start()

            def wait_a2(k):
                r = k * CH if isinstance(k, int) else pl.multiple_of(k * CH, CH)
                rcopy(xsend.at[pl.ds(r, CH), :], xrecv.at[pl.ds(r, CH), :],
                      ss.at[S_X], xr.at[k], xnb).wait_recv()

            def own(r, n):
                return (0, pl.ds(pl.multiple_of(own0 + r, 32), n), slice(None))

            def oth(r, n):
                return (0, pl.ds(pl.multiple_of(oth0 + r, 32), n), slice(None))

            def p1(i, c):
                wait_a2(2 * i)
                wait_a2(2 * i + 1)
                r = pl.multiple_of(i * 128, 128)
                v = _mlp(xrecv[pl.ds(r, 128), :], wbin[0], wbout[0]).astype(BF)
                a3[pl.ds(r, 128), :] = v
                pown[pl.ds(r, 128), :] = _mlp(v, wbin[1, :, pl.ds(0, HH)], wbout[1, pl.ds(0, HH), :])
                return c

            def fcopy():
                return rcopy(a3.at[pl.ds(0, FILL), :], yrecv.at[pl.ds(0, FILL), :],
                             ss.at[S_F], yr.at[NDIR], ynb)

            nfb = (FILL + 127) // 128
            with scope("s1_p1"):
                lax.fori_loop(0, nfb, p1, 0)
                fcopy().start()
                lax.fori_loop(nfb, N1, p1, 0)
            with scope("s1_wait_w3"):
                y_win(1).wait_recv()
                y_wout(1).wait_recv()

            def l3rem(r, n, pack=True):
                o = pown[pl.ds(r, n), :] + _mlp(
                    a3[pl.ds(r, n), :], wbin[1, :, pl.ds(HH, HH)], wbout[1, pl.ds(HH, HH), :])
                out[own(r, n)] = o
                if pack:
                    ysend[pl.ds(r, n), :] = o.astype(BF)

            def dcopy(j):
                r, n = DIR[j]
                return rcopy(ysend.at[pl.ds(r, n), :], yrecv.at[pl.ds(r, n), :],
                             ss.at[S_Y], yr.at[j], ynb)

            def rel_x(j):
                a, n, o = RELP[j]
                return rcopy(xrecv.at[pl.ds(RB + a, n), :], yrecv.at[pl.ds(o, n), :],
                             ss.at[S_RX], xr.at[NCH + j], xnb)

            def conv(r, n):
                out[oth(r, n)] = yrecv[pl.ds(r, n), :].astype(F32)

            with scope("s1_p2"):
                for j in range(ND2):
                    l3rem(*DIR[j])
                    dcopy(j).start()

            done = 0
            for b in range(N1, 16):
                with scope(f"s1_b{b}"):
                    r = b * 128
                    wait_a2(2 * b)
                    wait_a2(2 * b + 1)
                    upto = cfg["conv_at"].get(b, done)
                    for j in range(done, upto):
                        dcopy(j).wait_recv()
                    if b >= G0:
                        v = _mlp(xrecv[pl.ds(r, CH), :], wbin[0], wbout[0]).astype(BF)
                        v = jnp.concatenate([v, xrecv[pl.ds(r + CH, CH), :]], axis=0)
                    else:
                        v = _mlp(xrecv[pl.ds(r, 128), :], wbin[0], wbout[0]).astype(BF)
                    o = _mlp(v, wbin[1], wbout[1])
                    out[own(r, 128)] = o
                    ysend[pl.ds(r, 128), :] = o.astype(BF)
                    for j in range(done, upto):
                        conv(*DIR[j])
                    done = max(done, upto)
                    if b in RELB:
                        bi = RELB.index(b)
                        rcopy(ysend.at[pl.ds(r, 128), :], xrecv.at[pl.ds(bi * 128, 128), :],
                              ss.at[S_RX], xr.at[0 if b in REL1 else 1], xnb).start()
                    else:
                        for j in blk_msgs[b]:
                            dcopy(j).start()
            with scope("s1_fill"):
                fcopy().wait_recv()
                l3rem(0, FILL, pack=False)
                out[oth(0, FILL)] = _mlp(yrecv[pl.ds(0, FILL), :], wbin[1], wbout[1])
            with scope("s1_tail"):
                ev = []
                rem = 0
                for j in reversed(range(done, NDIR)):
                    ev.append((-rem, 0, j))
                    rem += DIR[j][1]
                rem = cfg.get("relay_early", 64)
                for j in reversed(range(NREL)):
                    ev.append((-rem, 1, j))
                    rem += RELP[j][1]
                ev.sort()
                for (_, kind, j) in ev:
                    if kind == 0:
                        dcopy(j).wait_recv()
                        conv(*DIR[j])
                    else:
                        rel_x(j).wait_recv()
                        conv(RELP[j][2], RELP[j][1])

        def rows(ref, n):
            return ref.at[pl.ds(0, n), :]

        with scope("s0_fin"):
            y_win(0).wait_send()
            y_wout(0).wait_send()

            @pl.when(mx == 0)
            def _():
                rcopy(ysend, yrecv, ss.at[S_Y], yr.at[0], ynb).wait_send()
                pltpu.make_async_copy(big, out.at[0], ss.at[S_Z]).wait()
                rcopy(xsend, xrecv, ss.at[S_X], xr.at[0], xnb).wait_send()
                if Z:
                    rcopy(rows(xrecv, Z), rows(xrecv, Z), ss.at[S_RY], yr.at[0], ynb).wait_send()
                    rcopy(rows(xrecv, Z), rows(yrecv, Z), ss.at[S_RX], xr.at[0], xnb).wait_send()

            @pl.when(mx == 1)
            def _():
                y_win(1).wait_send()
                y_wout(1).wait_send()
                for h in range(2):
                    x_win(h).wait_send()
                    x_wout(h).wait_send()
                rcopy(rows(xsend, FILL), rows(yrecv, FILL), ss.at[S_F], yr.at[0], ynb).wait_send()
                if Z:
                    rcopy(rows(ysend, Z), rows(xrecv, Z), ss.at[S_RX], xr.at[0], xnb).wait_send()
                rcopy(rows(ysend, NDROWS), rows(yrecv, NDROWS), ss.at[S_Y], yr.at[0], ynb).wait_send()

    def fn(x_padded, Win, Wout):
        return pl.pallas_call(
            body,
            out_shape=jax.ShapeDtypeStruct((1, NB, DM), F32),
            in_specs=[pl.BlockSpec(memory_space=pl.ANY)] * 3,
            out_specs=pl.BlockSpec(memory_space=pltpu.VMEM),
            scratch_shapes=[
                pltpu.VMEM((NB, DM), F32),
                pltpu.VMEM((HALF, DM), F32),
                pltpu.VMEM((512, DM), F32),
                pltpu.VMEM((2, DM, HH), F32),
                pltpu.VMEM((2, HH, DM), F32),
                pltpu.VMEM((3, DM, 2 * HH), BF),
                pltpu.VMEM((3, 2 * HH, DM), BF),
                pltpu.VMEM((HALF, DM), BF),
                pltpu.VMEM((HALF, DM), BF),
                pltpu.VMEM((HALF, DM), BF),
                pltpu.VMEM((HALF, DM), BF),
            ],
            compiler_params=pltpu.CompilerParams(
                collective_id=0, vmem_limit_bytes=48 * 1024 * 1024),
        )(x_padded, Win, Wout)

    return fn


_KERNEL_CFG = {}


def pallas_dist_pipemlp_pp2tp2_xy_b4096_d256_h512_kernel(x_padded, Win, Wout):
    return make(**_KERNEL_CFG)(x_padded, Win, Wout)
```

```python
import contextlib
import jax
import jax.numpy as jnp
from jax import lax
from jax.experimental import pallas as pl
from jax.experimental.pallas import tpu as pltpu

BF = jnp.bfloat16
F32 = jnp.float32
MESH = pl.DeviceIdType.MESH

NB = 4096
DM = 256
HH = 512
HALF = 2048
CH = 64
NCH = HALF // CH


def _mlp(a, win, wout):
    h = jnp.dot(a, win, preferred_element_type=F32)
    h = jnp.maximum(h, 0.0).astype(BF)
    return jnp.dot(h, wout, preferred_element_type=F32)


def _split(total, sizes, base=0):
    out, s, i = [], 0, 0
    while s < total:
        z = min(sizes[min(i, len(sizes) - 1)], total - s)
        out.append((base + s, z))
        s += z
        i += 1
    return out


DEFAULT = dict(
    fill=192,
    n1=6,
    p2=(128, 448),
    g0=8,
    rel1=(6, 7),
    rel2=(10,),
    kf=14,
    relp=64,
    last_split=(64, 32, 32),
    conv_at={8: 1, 12: 2, 13: 3, 14: 4, 15: 5},
    scopes=False,
)


def make(**kw):
    cfg = dict(DEFAULT)
    cfg.update(kw)
    FILL = cfg["fill"]
    N1 = cfg["n1"]
    G0 = cfg["g0"]
    KF = cfg["kf"]
    P1R = N1 * 128
    NE = cfg.get("ne", 6)
    assert FILL + sum(cfg["p2"]) == P1R
    REL1 = list(cfg["rel1"])
    REL2 = list(cfg["rel2"])
    RELB = REL1 + REL2
    Z = 128 * len(RELB)
    RELP = []
    for bi, b in enumerate(RELB):
        sizes = (cfg["relp"],)
        if bi == len(RELB) - 1:
            sizes = cfg.get("rel_last", (64, 32, 32))
        for (a, n) in _split(128, sizes):
            RELP.append((bi * 128 + a, n, b * 128 + a))
    NREL = len(RELP)
    NREL1 = sum(1 for p in RELP if p[0] < 128 * len(REL1))
    DIR = _split(P1R - FILL, cfg["p2"], FILL)
    ND2 = len(DIR)
    blk_msgs = {}
    for b in range(N1, 16):
        if b in RELB:
            continue
        parts = _split(128, cfg["last_split"], b * 128) if b == 15 else [(b * 128, 128)]
        blk_msgs[b] = list(range(len(DIR), len(DIR) + len(parts)))
        DIR += parts
    NDIR = len(DIR)
    NDROWS = sum(n for _, n in DIR)

    WINP = _split(DM, cfg.get("win_pieces", (32, 96, 128)))

    def scope(name):
        if cfg["scopes"]:
            return jax.named_scope(name)
        return contextlib.nullcontext()

    def body(x_hbm, win_hbm, wout_hbm, out,
             big, pown, zbuf, wfin, wfout, wbin, wbout,
             ysend, yrecv, xsend, xrecv):
        def scoped(ld, wr, yr, xr, ss):
            inner(x_hbm, win_hbm, wout_hbm, out, big, pown, zbuf, wfin, wfout, wbin, wbout,
                  ysend, yrecv, xsend, xrecv, ld, wr, yr, xr, ss)
        pl.run_scoped(
            scoped,
            pltpu.SemaphoreType.DMA((32,)),
            pltpu.SemaphoreType.DMA((8,)),
            pltpu.SemaphoreType.DMA((max(NCH + NREL, NDIR + 1),)),
            pltpu.SemaphoreType.DMA((NCH + NREL,)),
            pltpu.SemaphoreType.DMA((16,)),
        )

    def inner(x_hbm, win_hbm, wout_hbm, out,
              big, pown, zbuf, wfin, wfout, wbin, wbout,
              ysend, yrecv, xsend, xrecv,
              ld, wr, yr, xr, ss):
        mx = lax.axis_index("x")
        my = lax.axis_index("y")
        ynb = (mx, 1 - my)
        xnb = (1 - mx, my)
        own0 = my * HALF
        oth0 = (1 - my) * HALF
        bar = pltpu.get_barrier_semaphore()

        def rcopy(src, dst, ssem, rsem, dev):
            return pltpu.make_async_remote_copy(
                src_ref=src, dst_ref=dst, send_sem=ssem, recv_sem=rsem,
                device_id=dev, device_id_type=MESH)

        hb = [1 - mx, mx]
        NP = len(WINP)
        L_WO0, L_WI1, L_WO1, L_X = NP, NP + 1, NP + 2, NP + 3

        def ld_win(slot, r0, n, k):
            return pltpu.make_async_copy(
                win_hbm.at[hb[slot], pl.ds(r0, n), :], wfin.at[slot, pl.ds(r0, n), :], ld.at[k])

        def ld_wout(slot, k):
            return pltpu.make_async_copy(wout_hbm.at[hb[slot]], wfout.at[slot], ld.at[k])

        def cv_win(slot, r0, n):
            wbin[slot, pl.ds(r0, n), pl.ds(0, HH)] = wfin[slot, pl.ds(r0, n), :].astype(BF)

        def cv_wout(slot):
            wbout[slot, pl.ds(0, HH), :] = wfout[slot].astype(BF)

        def y_win(slot, r0=0, n=DM):
            return rcopy(wbin.at[slot, pl.ds(r0, n), pl.ds(0, HH)],
                         wbin.at[slot, pl.ds(r0, n), pl.ds(HH, HH)],
                         ss.at[2 * slot], wr.at[2 * slot], ynb)

        def y_wout(slot):
            return rcopy(wbout.at[slot, pl.ds(0, HH), :], wbout.at[slot, pl.ds(HH, HH), :],
                         ss.at[2 * slot + 1], wr.at[2 * slot + 1], ynb)

        def x_win(half, r0=0, n=DM):
            return rcopy(wbin.at[0, pl.ds(r0, n), pl.ds(half * HH, HH)],
                         wbin.at[2, pl.ds(r0, n), pl.ds(half * HH, HH)],
                         ss.at[4 + 2 * half], wr.at[4 + 2 * half], xnb)

        def x_wout(half):
            return rcopy(wbout.at[0, pl.ds(half * HH, HH), :], wbout.at[2, pl.ds(half * HH, HH), :],
                         ss.at[5 + 2 * half], wr.at[5 + 2 * half], xnb)

        S_Y, S_X, S_RY, S_RX, S_F, S_Z = 8, 9, 10, 11, 12, 13
        RB = 1024

        def xload(i):
            base = oth0 if i % 2 == 0 else own0
            off = pl.multiple_of(base + (i // 2) * 256, 256)
            return pltpu.make_async_copy(
                x_hbm.at[0, pl.ds(off, 256), :], big.at[pl.ds(i * 256, 256), :], ld.at[L_X + i // 2])

        with scope("s0_pro"):
            pl.semaphore_signal(bar, inc=1, device_id=ynb, device_id_type=MESH)
            ld_win(0, *WINP[0], 0).start()
            ld_win(0, *WINP[1], 1).start()

            @pl.when(mx == 0)
            def _():
                pl.semaphore_signal(bar, inc=1, device_id=xnb, device_id_type=MESH)
                ld_win(1, 0, DM, L_WI1).start()
                xload(0).start()
                xload(1).start()
                ld_wout(1, L_WO1).start()
                for j in range(2, NP):
                    ld_win(0, *WINP[j], j).start()
                xload(2).start()
                xload(3).start()
                ld_wout(0, L_WO0).start()
                for i in range(4, 16):
                    xload(i).start()

            @pl.when(mx == 1)
            def _():
                for j in range(2, NP):
                    ld_win(0, *WINP[j], j).start()
                ld_wout(0, L_WO0).start()
                ld_win(1, 0, DM, L_WI1).start()
                ld_wout(1, L_WO1).start()

            ld_win(0, *WINP[0], 0).wait()
            cv_win(0, *WINP[0])
            pl.semaphore_wait(bar, 1 + mx)
            y_win(0, *WINP[0]).start()
            ld_win(0, *WINP[1], 1).wait()
            cv_win(0, *WINP[1])
            y_win(0, *WINP[1]).start()

        @pl.when(mx == 0)
        def _stage0():
            with scope("s0_init"):
                ld_win(1, 0, DM, L_WI1).wait()
                cv_win(1, 0, DM)
                ld_wout(1, L_WO1).wait()
                cv_wout(1)

            def xwait(i):
                r = i * 512 if isinstance(i, int) else pl.multiple_of(i * 512, 512)
                pltpu.make_async_copy(
                    big.at[pl.ds(r, 512), :], big.at[pl.ds(r, 512), :], ld.at[L_X + i]).wait()

            def l0(row, n):
                a = big[pl.ds(row, n), :].astype(BF)
                return _mlp(a, wbin[1, :, pl.ds(0, HH)], wbout[1, pl.ds(0, HH), :])

            def psend(k):
                r = k * CH if isinstance(k, int) else pl.multiple_of(k * CH, CH)
                return rcopy(ysend.at[pl.ds(r, CH), :], yrecv.at[pl.ds(r, CH), :],
                             ss.at[S_Y], yr.at[k], ynb)

            def l0_blk(i):
                dyn = not isinstance(i, int)
                r = pl.multiple_of(i * 512, 512) if dyn else i * 512
                q = pl.multiple_of(i * 256, 256) if dyn else i * 256
                p = l0(r, 512)
                ysend[pl.ds(q, 256), :] = p[:256].astype(BF)
                pown[pl.ds(q, 256), :] = p[256:]

            with scope("s0_l0"):
                xwait(0)
                for j in range(2, NP):
                    ld_win(0, *WINP[j], j).wait()
                for j in range(2, NP):
                    cv_win(0, *WINP[j])
                    y_win(0, *WINP[j]).start()
                l0_blk(0)
                ld_wout(0, L_WO0).wait()
                xwait(1)
                cv_wout(0)
                y_wout(0).start()
                for k in range(4):
                    psend(k).start()

                def it(i, c):
                    l0_blk(i)
                    xwait(i + 1)
                    for q in range(4):
                        psend(i * 4 + q).start()
                    return c
                lax.fori_loop(1, NE, it, 0)
                for i in range(NE + 1, 8):
                    xwait(i)
                zbuf[...] = jnp.zeros_like(zbuf)
                for i in range(NB // 512):
                    pltpu.make_async_copy(zbuf, out.at[0, pl.ds(i * 512, 512), :], ss.at[S_Z]).start()

            with scope("s0_wait_w1"):
                y_win(0).wait_recv()
                y_wout(0).wait_recv()
                x_win(0).wait_recv()

            def chunk(k, g3, extra=None):
                r = pl.multiple_of(k * CH, CH)
                psend(k).wait_recv()
                a = (pown[pl.ds(r, CH), :] + yrecv[pl.ds(r, CH), :].astype(F32)).astype(BF)
                a = _mlp(a, wbin[0], wbout[0]).astype(BF)
                if g3:
                    a = _mlp(a, wbin[2], wbout[2]).astype(BF)
                xsend[pl.ds(r, CH), :] = a
                if extra is not None:
                    extra()
                rcopy(xsend.at[pl.ds(r, CH), :], xrecv.at[pl.ds(r, CH), :],
                      ss.at[S_X], xr.at[k], xnb).start()

            def pair_late(j, c):
                chunk(2 * j, False)
                kk = NE * 4 + j
                q = pl.multiple_of(kk * CH, CH)
                rb = pl.multiple_of((kk // 4) * 512 + (kk % 4) * CH, CH)

                def extra():
                    a = jnp.concatenate(
                        [big[pl.ds(rb, CH), :], big[pl.ds(pl.multiple_of(rb + 256, CH), CH), :]],
                        axis=0).astype(BF)
                    p = _mlp(a, wbin[1, :, pl.ds(0, HH)], wbout[1, pl.ds(0, HH), :])
                    ysend[pl.ds(q, CH), :] = p[:CH].astype(BF)
                    pown[pl.ds(q, CH), :] = p[CH:]
                chunk(2 * j + 1, False, extra)
                psend(kk).start()
                return c

            def pair_plain(j, c):
                chunk(2 * j, False)
                chunk(2 * j + 1, False)
                return c

            def pair_g3(j, c):
                chunk(2 * j, False)
                chunk(2 * j + 1, True)
                return c

            def rel_in(lo, hi, sem):
                return rcopy(ysend.at[pl.ds(lo, hi - lo), :], xrecv.at[pl.ds(lo, hi - lo), :],
                             ss.at[S_RX], xr.at[sem], xnb)

            def rel_y(j):
                a, n, _ = RELP[j]
                return rcopy(xrecv.at[pl.ds(a, n), :], xrecv.at[pl.ds(RB + a, n), :],
                             ss.at[S_RY], yr.at[NCH + j], ynb)

            def rel_x(j):
                a, n, o = RELP[j]
                return rcopy(xrecv.at[pl.ds(RB + a, n), :], yrecv.at[pl.ds(o, n), :],
                             ss.at[S_RX], xr.at[NCH + j], xnb)

            with scope("s0_p2a"):
                NL = (8 - NE) * 4
                lax.fori_loop(0, NL, pair_late, 0)
                if G0 > NL:
                    lax.fori_loop(NL, G0, pair_plain, 0)
            with scope("s0_wait_w2"):
                x_wout(0).wait_recv()
                x_win(1).wait_recv()
                x_wout(1).wait_recv()
            with scope("s0_p2b"):
                lax.fori_loop(G0, KF, pair_g3, 0)
            with scope("s0_relay1"):
                if REL1:
                    rel_in(0, 128 * len(REL1), 0).wait_recv()
                    for j in range(NREL1):
                        rel_y(j).start()
            with scope("s0_p2c"):
                lax.fori_loop(KF, 16, pair_g3, 0)
            with scope("s0_relay2"):
                if REL2:
                    rel_in(128 * len(REL1), Z, 1).wait_recv()
                    for j in range(NREL1, NREL):
                        rel_y(j).start()
                for j in range(NREL):
                    rel_y(j).wait_recv()
                    rel_x(j).start()

        @pl.when(mx == 1)
        def _stage1():
            a3 = xsend
            with scope("s1_init"):
                x_win(0, 0, WINP[2][0]).start()
                for j in range(2, NP):
                    ld_win(0, *WINP[j], j).wait()
                    cv_win(0, *WINP[j])
                    y_win(0, *WINP[j]).start()
                    x_win(0, *WINP[j]).start()
                ld_wout(0, L_WO0).wait()
                cv_wout(0)
                y_wout(0).start()
                x_wout(0).start()
                ld_win(1, 0, DM, L_WI1).wait()
                cv_win(1, 0, DM)
                y_win(1).start()
                ld_wout(1, L_WO1).wait()
                cv_wout(1)
                y_wout(1).start()
            with scope("s1_wait_w2"):
                y_win(0).wait_recv()
                x_win(1).start()
                y_wout(0).wait_recv()
                x_wout(1).start()

            def wait_a2(k):
                r = k * CH if isinstance(k, int) else pl.multiple_of(k * CH, CH)
                rcopy(xsend.at[pl.ds(r, CH), :], xrecv.at[pl.ds(r, CH), :],
                      ss.at[S_X], xr.at[k], xnb).wait_recv()

            def own(r, n):
                return (0, pl.ds(pl.multiple_of(own0 + r, 32), n), slice(None))

            def oth(r, n):
                return (0, pl.ds(pl.multiple_of(oth0 + r, 32), n), slice(None))

            def p1(i, c):
                wait_a2(2 * i)
                wait_a2(2 * i + 1)
                r = pl.multiple_of(i * 128, 128)
                v = _mlp(xrecv[pl.ds(r, 128), :], wbin[0], wbout[0]).astype(BF)
                a3[pl.ds(r, 128), :] = v
                pown[pl.ds(r, 128), :] = _mlp(v, wbin[1, :, pl.ds(0, HH)], wbout[1, pl.ds(0, HH), :])
                return c

            def fcopy():
                return rcopy(a3.at[pl.ds(0, FILL), :], yrecv.at[pl.ds(0, FILL), :],
                             ss.at[S_F], yr.at[NDIR], ynb)

            nfb = (FILL + 127) // 128
            with scope("s1_p1"):
                lax.fori_loop(0, nfb, p1, 0)
                fcopy().start()
                lax.fori_loop(nfb, N1, p1, 0)
            with scope("s1_wait_w3"):
                y_win(1).wait_recv()
                y_wout(1).wait_recv()

            def l3rem(r, n, pack=True):
                o = pown[pl.ds(r, n), :] + _mlp(
                    a3[pl.ds(r, n), :], wbin[1, :, pl.ds(HH, HH)], wbout[1, pl.ds(HH, HH), :])
                out[own(r, n)] = o
                if pack:
                    ysend[pl.ds(r, n), :] = o.astype(BF)

            def dcopy(j):
                r, n = DIR[j]
                return rcopy(ysend.at[pl.ds(r, n), :], yrecv.at[pl.ds(r, n), :],
                             ss.at[S_Y], yr.at[j], ynb)

            def rel_x(j):
                a, n, o = RELP[j]
                return rcopy(xrecv.at[pl.ds(RB + a, n), :], yrecv.at[pl.ds(o, n), :],
                             ss.at[S_RX], xr.at[NCH + j], xnb)

            def conv(r, n):
                out[oth(r, n)] = yrecv[pl.ds(r, n), :].astype(F32)

            with scope("s1_p2"):
                for j in range(ND2):
                    l3rem(*DIR[j])
                    dcopy(j).start()

            done = 0
            for b in range(N1, 16):
                with scope(f"s1_b{b}"):
                    r = b * 128
                    wait_a2(2 * b)
                    wait_a2(2 * b + 1)
                    upto = cfg["conv_at"].get(b, done)
                    for j in range(done, upto):
                        dcopy(j).wait_recv()
                    if b >= G0:
                        v = _mlp(xrecv[pl.ds(r, CH), :], wbin[0], wbout[0]).astype(BF)
                        v = jnp.concatenate([v, xrecv[pl.ds(r + CH, CH), :]], axis=0)
                    else:
                        v = _mlp(xrecv[pl.ds(r, 128), :], wbin[0], wbout[0]).astype(BF)
                    o = _mlp(v, wbin[1], wbout[1])
                    out[own(r, 128)] = o
                    ysend[pl.ds(r, 128), :] = o.astype(BF)
                    for j in range(done, upto):
                        conv(*DIR[j])
                    done = max(done, upto)
                    if b in RELB:
                        bi = RELB.index(b)
                        rcopy(ysend.at[pl.ds(r, 128), :], xrecv.at[pl.ds(bi * 128, 128), :],
                              ss.at[S_RX], xr.at[0 if b in REL1 else 1], xnb).start()
                    else:
                        for j in blk_msgs[b]:
                            dcopy(j).start()
            with scope("s1_fill"):
                fcopy().wait_recv()
                l3rem(0, FILL, pack=False)
                out[oth(0, FILL)] = _mlp(yrecv[pl.ds(0, FILL), :], wbin[1], wbout[1])
            with scope("s1_tail"):
                ev = []
                rem = 0
                for j in reversed(range(done, NDIR)):
                    ev.append((-rem, 0, j))
                    rem += DIR[j][1]
                rem = cfg.get("relay_early", 64)
                for j in reversed(range(NREL)):
                    ev.append((-rem, 1, j))
                    rem += RELP[j][1]
                ev.sort()
                for (_, kind, j) in ev:
                    if kind == 0:
                        dcopy(j).wait_recv()
                        conv(*DIR[j])
                    else:
                        rel_x(j).wait_recv()
                        conv(RELP[j][2], RELP[j][1])

        def rows(ref, n):
            return ref.at[pl.ds(0, n), :]

        with scope("s0_fin"):
            y_win(0).wait_send()
            y_wout(0).wait_send()

            @pl.when(mx == 0)
            def _():
                rcopy(ysend, yrecv, ss.at[S_Y], yr.at[0], ynb).wait_send()
                pltpu.make_async_copy(big, out.at[0], ss.at[S_Z]).wait()
                rcopy(xsend, xrecv, ss.at[S_X], xr.at[0], xnb).wait_send()
                if Z:
                    rcopy(rows(xrecv, Z), rows(xrecv, Z), ss.at[S_RY], yr.at[0], ynb).wait_send()
                    rcopy(rows(xrecv, Z), rows(yrecv, Z), ss.at[S_RX], xr.at[0], xnb).wait_send()

            @pl.when(mx == 1)
            def _():
                y_win(1).wait_send()
                y_wout(1).wait_send()
                for h in range(2):
                    x_win(h).wait_send()
                    x_wout(h).wait_send()
                rcopy(rows(xsend, FILL), rows(yrecv, FILL), ss.at[S_F], yr.at[0], ynb).wait_send()
                if Z:
                    rcopy(rows(ysend, Z), rows(xrecv, Z), ss.at[S_RX], xr.at[0], xnb).wait_send()
                rcopy(rows(ysend, NDROWS), rows(yrecv, NDROWS), ss.at[S_Y], yr.at[0], ynb).wait_send()

    def fn(x_padded, Win, Wout):
        return pl.pallas_call(
            body,
            out_shape=jax.ShapeDtypeStruct((1, NB, DM), F32),
            in_specs=[pl.BlockSpec(memory_space=pl.ANY)] * 3,
            out_specs=pl.BlockSpec(memory_space=pltpu.VMEM),
            scratch_shapes=[
                pltpu.VMEM((NB, DM), F32),
                pltpu.VMEM((HALF, DM), F32),
                pltpu.VMEM((512, DM), F32),
                pltpu.VMEM((2, DM, HH), F32),
                pltpu.VMEM((2, HH, DM), F32),
                pltpu.VMEM((3, DM, 2 * HH), BF),
                pltpu.VMEM((3, 2 * HH, DM), BF),
                pltpu.VMEM((HALF, DM), BF),
                pltpu.VMEM((HALF, DM), BF),
                pltpu.VMEM((HALF, DM), BF),
                pltpu.VMEM((HALF, DM), BF),
            ],
            compiler_params=pltpu.CompilerParams(
                collective_id=0, vmem_limit_bytes=48 * 1024 * 1024),
        )(x_padded, Win, Wout)

    return fn


_KERNEL_CFG = {}


def pallas_dist_pipemlp_pp2tp2_xy_b4096_d256_h512_kernel(x_padded, Win, Wout):
    return make(**_KERNEL_CFG)(x_padded, Win, Wout)
```

```python
import contextlib
import jax
import jax.numpy as jnp
from jax import lax
from jax.experimental import pallas as pl
from jax.experimental.pallas import tpu as pltpu

BF = jnp.bfloat16
F32 = jnp.float32
MESH = pl.DeviceIdType.MESH

NB = 4096
DM = 256
HH = 512
HALF = 2048
CH = 64
NCH = HALF // CH


def _mlp(a, win, wout):
    h = jnp.dot(a, win, preferred_element_type=F32)
    h = jnp.maximum(h, 0.0).astype(BF)
    return jnp.dot(h, wout, preferred_element_type=F32)


def _split(total, sizes, base=0):
    out, s, i = [], 0, 0
    while s < total:
        z = min(sizes[min(i, len(sizes) - 1)], total - s)
        out.append((base + s, z))
        s += z
        i += 1
    return out


DEFAULT = dict(
    fill=160,
    na=2,
    n1=6,
    p2=(96, 384, 128),
    g0=8,
    rel=(((1152, 128),), ((1280, 128),), ((1408, 64),), ((1536, 80),)),
    kf=15,
    relp=64,
    order=("i1", "x0", "i2", "x1", "i3", "x2", "x3", "x4", "x5", "x6"),
    last_split=(64, 32, 32),
    conv_at={8: 1, 11: 2, 12: 3, 13: 4, 14: 5, 15: 6},
    scopes=False,
)


def make(**kw):
    cfg = dict(DEFAULT)
    cfg.update(kw)
    FILL = cfg["fill"]
    N1 = cfg["n1"]
    G0 = cfg["g0"]
    KF = cfg["kf"]
    P1R = N1 * 128
    NE = cfg.get("ne", 6)
    assert FILL + sum(cfg["p2"]) == P1R
    RELP = []
    GRP = []
    blk_rel = {}
    Z = 0
    for g, grp in enumerate(cfg["rel"]):
        lo = Z
        idx = []
        for (r, n) in grp:
            assert r % 128 == 0 and n <= 128
            blk_rel[r // 128] = (Z, n, g)
            for (a, m) in _split(n, (cfg["relp"],)):
                idx.append(len(RELP))
                RELP.append((Z + a, m, r + a))
            Z += n
        GRP.append((lo, Z, idx))
    NREL = len(RELP)
    DIR = _split(P1R - FILL, cfg["p2"], FILL)
    ND2 = len(DIR)
    blk_msgs = {}
    for b in range(N1, 16):
        skip = blk_rel[b][1] if b in blk_rel else 0
        if skip == 128:
            parts = []
        elif b == 15:
            parts = _split(128 - skip, cfg["last_split"], b * 128 + skip)
        else:
            parts = [(b * 128 + skip, 128 - skip)]
        blk_msgs[b] = list(range(len(DIR), len(DIR) + len(parts)))
        DIR += parts
    NDIR = len(DIR)
    NDROWS = sum(n for _, n in DIR)

    DONE = max(cfg["conv_at"].values())
    EV = []
    rem = 0
    for j in reversed(range(DONE, NDIR)):
        EV.append((-rem, 0, j))
        rem += DIR[j][1]
    rem = cfg.get("relay_early", 32)
    for j in reversed(range(NREL)):
        EV.append((-rem, 1, j))
        rem += RELP[j][1]
    EV.sort()
    NLAST = cfg.get("nlast", 4)

    WINP = _split(DM, cfg.get("win_pieces", (16, 48, 96, 96)))

    def scope(name):
        if cfg["scopes"]:
            return jax.named_scope(name)
        return contextlib.nullcontext()

    def body(x_hbm, win_hbm, wout_hbm, out,
             big, pown, zbuf, wfin, wfout, wbin, wbout,
             ysend, yrecv, xsend, xrecv, hbuf):
        def scoped(ld, wr, yr, xr, ss):
            inner(x_hbm, win_hbm, wout_hbm, out, big, pown, zbuf, wfin, wfout, wbin, wbout,
                  ysend, yrecv, xsend, xrecv, hbuf, ld, wr, yr, xr, ss)
        pl.run_scoped(
            scoped,
            pltpu.SemaphoreType.DMA((32,)),
            pltpu.SemaphoreType.DMA((8,)),
            pltpu.SemaphoreType.DMA((max(NCH + NREL, NDIR + 1),)),
            pltpu.SemaphoreType.DMA((NCH + NREL,)),
            pltpu.SemaphoreType.DMA((16,)),
        )

    def inner(x_hbm, win_hbm, wout_hbm, out,
              big, pown, zbuf, wfin, wfout, wbin, wbout,
              ysend, yrecv, xsend, xrecv, hbuf,
              ld, wr, yr, xr, ss):
        mx = lax.axis_index("x")
        my = lax.axis_index("y")
        ynb = (mx, 1 - my)
        xnb = (1 - mx, my)
        own0 = my * HALF
        oth0 = (1 - my) * HALF
        bar = pltpu.get_barrier_semaphore()

        def rcopy(src, dst, ssem, rsem, dev):
            return pltpu.make_async_remote_copy(
                src_ref=src, dst_ref=dst, send_sem=ssem, recv_sem=rsem,
                device_id=dev, device_id_type=MESH)

        hb = [1 - mx, mx]
        NP = len(WINP)
        NPRO = cfg.get("npro", 3)
        L_WO0, L_WI1, L_WO1, L_X = NP, NP + 1, NP + 2, NP + 3

        def ld_win(slot, r0, n, k):
            return pltpu.make_async_copy(
                win_hbm.at[hb[slot], pl.ds(r0, n), :], wfin.at[slot, pl.ds(r0, n), :], ld.at[k])

        def ld_wout(slot, k):
            return pltpu.make_async_copy(wout_hbm.at[hb[slot]], wfout.at[slot], ld.at[k])

        def cv_win(slot, r0, n):
            wbin[slot, pl.ds(r0, n), pl.ds(0, HH)] = wfin[slot, pl.ds(r0, n), :].astype(BF)

        def cv_wout(slot):
            wbout[slot, pl.ds(0, HH), :] = wfout[slot].astype(BF)

        def y_win(slot, r0=0, n=DM):
            return rcopy(wbin.at[slot, pl.ds(r0, n), pl.ds(0, HH)],
                         wbin.at[slot, pl.ds(r0, n), pl.ds(HH, HH)],
                         ss.at[2 * slot], wr.at[2 * slot], ynb)

        def y_wout(slot):
            return rcopy(wbout.at[slot, pl.ds(0, HH), :], wbout.at[slot, pl.ds(HH, HH), :],
                         ss.at[2 * slot + 1], wr.at[2 * slot + 1], ynb)

        def x_win(half, r0=0, n=DM):
            return rcopy(wbin.at[0, pl.ds(r0, n), pl.ds(half * HH, HH)],
                         wbin.at[2, pl.ds(r0, n), pl.ds(half * HH, HH)],
                         ss.at[4 + 2 * half], wr.at[4 + 2 * half], xnb)

        def x_wout(half):
            return rcopy(wbout.at[0, pl.ds(half * HH, HH), :], wbout.at[2, pl.ds(half * HH, HH), :],
                         ss.at[5 + 2 * half], wr.at[5 + 2 * half], xnb)

        S_Y, S_X, S_RY, S_RX, S_F, S_Z = 8, 9, 10, 11, 12, 13
        RB = 1024

        def xload(i):
            base = oth0 if i % 2 == 0 else own0
            off = pl.multiple_of(base + (i // 2) * 256, 256)
            return pltpu.make_async_copy(
                x_hbm.at[0, pl.ds(off, 256), :], big.at[pl.ds(i * 256, 256), :], ld.at[L_X + i // 2])

        def rows(ref, n):
            return ref.at[pl.ds(0, n), :]

        def oth(r, n):
            return (0, pl.ds(pl.multiple_of(oth0 + r, 16), n), slice(None))

        def dcopy(j):
            r, n = DIR[j]
            return rcopy(ysend.at[pl.ds(r, n), :], yrecv.at[pl.ds(r, n), :],
                         ss.at[S_Y], yr.at[j], ynb)

        def rel_x(j):
            a, n, o = RELP[j]
            return rcopy(xrecv.at[pl.ds(RB + a, n), :], yrecv.at[pl.ds(o, n), :],
                         ss.at[S_RX], xr.at[NCH + j], xnb)

        def conv(r, n):
            out[oth(r, n)] = yrecv[pl.ds(r, n), :].astype(F32)

        def tail_ev(e):
            _, kind, j = e
            with scope(f"s1_e{'dr'[kind]}{j}"):
                if kind == 0:
                    dcopy(j).wait_recv()
                    conv(*DIR[j])
                else:
                    rel_x(j).wait_recv()
                    conv(RELP[j][2], RELP[j][1])

        def rest_loads():
            @pl.when(mx == 0)
            def _():
                ld_win(1, 0, DM, L_WI1).start()
                xload(0).start()
                xload(1).start()
                ld_wout(1, L_WO1).start()
                for j in range(NPRO, NP):
                    ld_win(0, *WINP[j], j).start()
                xload(2).start()
                xload(3).start()
                ld_wout(0, L_WO0).start()
                for i in range(4, 16):
                    xload(i).start()

            @pl.when(mx == 1)
            def _():
                for j in range(NPRO, NP):
                    ld_win(0, *WINP[j], j).start()
                ld_wout(0, L_WO0).start()
                ld_win(1, 0, DM, L_WI1).start()
                ld_wout(1, L_WO1).start()

        PRO = cfg.get("pro", 0)
        with scope("s0_pro"):
            ld_win(0, *WINP[0], 0).start()
            pl.semaphore_signal(bar, inc=1, device_id=ynb, device_id_type=MESH)

            @pl.when(mx == 0)
            def _():
                pl.semaphore_signal(bar, inc=1, device_id=xnb, device_id_type=MESH)
            if PRO == 2:
                pl.delay(cfg.get("dly", 100))
            for j in range(1, NPRO):
                ld_win(0, *WINP[j], j).start()
            if PRO in (0, 2):
                rest_loads()
        with scope("s0_pa"):
            ld_win(0, *WINP[0], 0).wait()
            cv_win(0, *WINP[0])
            if PRO == 3:
                rest_loads()
        with scope("s0_pb"):
            if PRO == 1:
                @pl.when(my == 0)
                def _():
                    rest_loads()
            pl.semaphore_wait(bar, 1 + mx)
            y_win(0, *WINP[0]).start()
            if PRO == 1:
                @pl.when(my == 1)
                def _():
                    rest_loads()
        with scope("s0_pc"):
            for j in range(1, NPRO):
                ld_win(0, *WINP[j], j).wait()
                cv_win(0, *WINP[j])
                y_win(0, *WINP[j]).start()

        @pl.when(mx == 0)
        def _stage0():
            with scope("s0_init"):
                ld_win(1, 0, DM, L_WI1).wait()
                cv_win(1, 0, DM)
                ld_wout(1, L_WO1).wait()
                cv_wout(1)

            def xwait(i):
                r = i * 512 if isinstance(i, int) else pl.multiple_of(i * 512, 512)
                pltpu.make_async_copy(
                    big.at[pl.ds(r, 512), :], big.at[pl.ds(r, 512), :], ld.at[L_X + i]).wait()

            def l0(row, n):
                a = big[pl.ds(row, n), :].astype(BF)
                return _mlp(a, wbin[1, :, pl.ds(0, HH)], wbout[1, pl.ds(0, HH), :])

            def psend(k):
                r = k * CH if isinstance(k, int) else pl.multiple_of(k * CH, CH)
                return rcopy(ysend.at[pl.ds(r, CH), :], yrecv.at[pl.ds(r, CH), :],
                             ss.at[S_Y], yr.at[k], ynb)

            def l0_blk(i):
                dyn = not isinstance(i, int)
                r = pl.multiple_of(i * 512, 512) if dyn else i * 512
                q = pl.multiple_of(i * 256, 256) if dyn else i * 256
                p = l0(r, 512)
                ysend[pl.ds(q, 256), :] = p[:256].astype(BF)
                pown[pl.ds(q, 256), :] = p[256:]

            with scope("s0_l0"):
                xwait(0)
                for j in range(NPRO, NP):
                    ld_win(0, *WINP[j], j).wait()
                for j in range(NPRO, NP):
                    cv_win(0, *WINP[j])
                    y_win(0, *WINP[j]).start()
                l0_blk(0)
                ld_wout(0, L_WO0).wait()
                xwait(1)
                cv_wout(0)
                y_wout(0).start()
                for k in range(4):
                    psend(k).start()

                def it(i, c):
                    l0_blk(i)
                    xwait(i + 1)
                    for q in range(4):
                        psend(i * 4 + q).start()
                    return c
                lax.fori_loop(1, NE, it, 0)
                for i in range(NE + 1, 8):
                    xwait(i)
                zbuf[...] = jnp.zeros_like(zbuf)
                for i in range(NB // 512):
                    pltpu.make_async_copy(zbuf, out.at[0, pl.ds(i * 512, 512), :], ss.at[S_Z]).start()

            with scope("s0_wait_w1"):
                y_win(0).wait_recv()
                y_wout(0).wait_recv()
                x_win(0).wait_recv()

            def chunk(k, g3, extra=None):
                r = pl.multiple_of(k * CH, CH)
                psend(k).wait_recv()
                a = (pown[pl.ds(r, CH), :] + yrecv[pl.ds(r, CH), :].astype(F32)).astype(BF)
                a = _mlp(a, wbin[0], wbout[0]).astype(BF)
                if g3:
                    a = _mlp(a, wbin[2], wbout[2]).astype(BF)
                xsend[pl.ds(r, CH), :] = a
                if extra is not None:
                    extra()
                rcopy(xsend.at[pl.ds(r, CH), :], xrecv.at[pl.ds(r, CH), :],
                      ss.at[S_X], xr.at[k], xnb).start()

            def pair_late(j, c):
                chunk(2 * j, False)
                kk = NE * 4 + j
                q = pl.multiple_of(kk * CH, CH)
                rb = pl.multiple_of((kk // 4) * 512 + (kk % 4) * CH, CH)

                def extra():
                    a = jnp.concatenate(
                        [big[pl.ds(rb, CH), :], big[pl.ds(pl.multiple_of(rb + 256, CH), CH), :]],
                        axis=0).astype(BF)
                    p = _mlp(a, wbin[1, :, pl.ds(0, HH)], wbout[1, pl.ds(0, HH), :])
                    ysend[pl.ds(q, CH), :] = p[:CH].astype(BF)
                    pown[pl.ds(q, CH), :] = p[CH:]
                chunk(2 * j + 1, False, extra)
                psend(kk).start()
                return c

            def pair_plain(j, c):
                chunk(2 * j, False)
                chunk(2 * j + 1, False)
                return c

            def pair_g3(j, c):
                chunk(2 * j, False)
                chunk(2 * j + 1, True)
                return c

            def rel_in(lo, hi, sem):
                return rcopy(ysend.at[pl.ds(lo, hi - lo), :], xrecv.at[pl.ds(lo, hi - lo), :],
                             ss.at[S_RX], xr.at[sem], xnb)

            def rel_y(j):
                a, n, _ = RELP[j]
                return rcopy(xrecv.at[pl.ds(a, n), :], xrecv.at[pl.ds(RB + a, n), :],
                             ss.at[S_RY], yr.at[NCH + j], ynb)

            with scope("s0_p2a"):
                NL = (8 - NE) * 4
                lax.fori_loop(0, NL, pair_late, 0)
                if G0 > NL:
                    lax.fori_loop(NL, G0, pair_plain, 0)
            with scope("s0_wait_w2"):
                x_wout(0).wait_recv()
                x_win(1).wait_recv()
                x_wout(1).wait_recv()
            with scope("s0_p2b"):
                lax.fori_loop(G0, KF, pair_g3, 0)
            def fwd_y(g):
                lo, hi, idx = GRP[g]
                rel_in(lo, hi, g).wait_recv()
                for j in idx:
                    rel_y(j).start()

            with scope("s0_relay1"):
                fwd_y(0)
            with scope("s0_p2c"):
                if KF < 16:
                    lax.fori_loop(KF, 16, pair_g3, 0)
            assert sorted(cfg["order"]) == sorted(
                [f"i{g}" for g in range(1, len(GRP))] + [f"x{j}" for j in range(NREL)])
            for ev in cfg["order"]:
                with scope("s0_" + ev):
                    j = int(ev[1:])
                    if ev[0] == "i":
                        fwd_y(j)
                    else:
                        rel_y(j).wait_recv()
                        rel_x(j).start()

        @pl.when(mx == 1)
        def _stage1():
            a3 = xsend
            with scope("s1_init"):
                x_win(0, 0, WINP[NPRO][0]).start()
                for j in range(NPRO, NP):
                    ld_win(0, *WINP[j], j).wait()
                    cv_win(0, *WINP[j])
                    y_win(0, *WINP[j]).start()
                    x_win(0, *WINP[j]).start()
                ld_wout(0, L_WO0).wait()
                cv_wout(0)
                y_wout(0).start()
                x_wout(0).start()
                ld_win(1, 0, DM, L_WI1).wait()
                cv_win(1, 0, DM)
                y_win(1).start()
                ld_wout(1, L_WO1).wait()
                cv_wout(1)
                y_wout(1).start()
            with scope("s1_wait_w2"):
                y_win(0).wait_recv()
                x_win(1).start()
                y_wout(0).wait_recv()
                x_wout(1).start()

            def wait_a2(k):
                r = k * CH if isinstance(k, int) else pl.multiple_of(k * CH, CH)
                rcopy(xsend.at[pl.ds(r, CH), :], xrecv.at[pl.ds(r, CH), :],
                      ss.at[S_X], xr.at[k], xnb).wait_recv()

            def own(r, n):
                return (0, pl.ds(pl.multiple_of(own0 + r, 16), n), slice(None))

            def p1(i, c):
                wait_a2(2 * i)
                wait_a2(2 * i + 1)
                r = pl.multiple_of(i * 128, 128)
                v = _mlp(xrecv[pl.ds(r, 128), :], wbin[0], wbout[0]).astype(BF)
                a3[pl.ds(r, 128), :] = v
                pown[pl.ds(r, 128), :] = _mlp(v, wbin[1, :, pl.ds(0, HH)], wbout[1, pl.ds(0, HH), :])
                return c

            def fcopy():
                return rcopy(a3.at[pl.ds(0, FILL), :], yrecv.at[pl.ds(0, FILL), :],
                             ss.at[S_F], yr.at[NDIR], ynb)

            W3I_L = (1, slice(None), pl.ds(0, HH))
            W3I_R = (1, slice(None), pl.ds(HH, HH))
            W3O_L = (1, pl.ds(0, HH), slice(None))
            W3O_R = (1, pl.ds(HH, HH), slice(None))

            def relu_mm(a, w):
                return jnp.maximum(jnp.dot(a, w, preferred_element_type=F32), 0.0).astype(BF)

            def p1h(i, back=0):
                wait_a2(2 * i)
                wait_a2(2 * i + 1)
                dyn = not isinstance(i, int)
                r = pl.multiple_of(i * 128, 128) if dyn else i * 128
                v = _mlp(xrecv[pl.ds(r, 128), :], wbin[0], wbout[0]).astype(BF)
                if back:
                    pown[pl.ds(r, 128), :] = _mlp(v, wbin[W3I_L], wbout[W3O_L])
                    vv = jnp.concatenate([a3[pl.ds(r - back, back), :], v], axis=0)
                    hbuf[pl.ds(r - back, 128 + back), :] = relu_mm(vv, wbin[W3I_R])
                else:
                    h = relu_mm(v, wbin[1])
                    hbuf[pl.ds(r, 128), :] = h[:, HH:]
                    pown[pl.ds(r, 128), :] = jnp.dot(h[:, :HH], wbout[W3O_L], preferred_element_type=F32)

            def l3rem(r, n, pack=True):
                o = pown[pl.ds(r, n), :] + _mlp(a3[pl.ds(r, n), :], wbin[W3I_R], wbout[W3O_R])
                out[own(r, n)] = o
                if pack:
                    ysend[pl.ds(r, n), :] = o.astype(BF)

            def orem(r, n):
                o = pown[pl.ds(r, n), :] + jnp.dot(
                    hbuf[pl.ds(r, n), :], wbout[W3O_R], preferred_element_type=F32)
                out[own(r, n)] = o
                ysend[pl.ds(r, n), :] = o.astype(BF)

            NA = cfg["na"]
            assert FILL <= NA * 128
            with scope("s1_p1a"):
                lax.fori_loop(0, NA, p1, 0)
                fcopy().start()
            with scope("s1_wait_w3i"):
                y_win(1).wait_recv()
            with scope("s1_p1b"):
                p1h(NA, NA * 128 - FILL)

                def it(i, c):
                    p1h(i)
                    return c
                lax.fori_loop(NA + 1, N1 - 1, it, 0)
            with scope("s1_p1c"):
                rl = (N1 - 1) * 128
                wait_a2(2 * N1 - 2)
                wait_a2(2 * N1 - 1)
                a3[pl.ds(rl, 128), :] = _mlp(xrecv[pl.ds(rl, 128), :], wbin[0], wbout[0]).astype(BF)
            with scope("s1_wait_w3"):
                y_wout(1).wait_recv()
            with scope("s1_p2"):
                for j in range(ND2 - 1):
                    orem(*DIR[j])
                    dcopy(j).start()
                assert DIR[ND2 - 1] == (rl, 128)
                o = _mlp(a3[pl.ds(rl, 128), :], wbin[1], wbout[1])
                out[own(rl, 128)] = o
                ysend[pl.ds(rl, 128), :] = o.astype(BF)
                dcopy(ND2 - 1).start()

            done = 0
            for b in range(N1, 16):
                with scope(f"s1_b{b}"):
                    r = b * 128
                    wait_a2(2 * b)
                    wait_a2(2 * b + 1)
                    upto = cfg["conv_at"].get(b, done)
                    for j in range(done, upto):
                        dcopy(j).wait_recv()
                    if b >= G0:
                        v = _mlp(xrecv[pl.ds(r, CH), :], wbin[0], wbout[0]).astype(BF)
                        v = jnp.concatenate([v, xrecv[pl.ds(r + CH, CH), :]], axis=0)
                    else:
                        v = _mlp(xrecv[pl.ds(r, 128), :], wbin[0], wbout[0]).astype(BF)
                    o = _mlp(v, wbin[1], wbout[1])
                    out[own(r, 128)] = o
                    ysend[pl.ds(r, 128), :] = o.astype(BF)
                    for j in range(done, upto):
                        conv(*DIR[j])
                    done = max(done, upto)
                    for j in blk_msgs[b]:
                        dcopy(j).start()
                    if b in blk_rel:
                        z0, zn, g = blk_rel[b]
                        rcopy(ysend.at[pl.ds(r, zn), :], xrecv.at[pl.ds(z0, zn), :],
                              ss.at[S_RX], xr.at[g], xnb).start()
            with scope("s1_fill"):
                fcopy().wait_recv()
                l3rem(0, FILL, pack=False)
                out[oth(0, FILL)] = _mlp(yrecv[pl.ds(0, FILL), :], wbin[1], wbout[1])
            with scope("s1_tail"):
                assert done == DONE
                for e in EV[:len(EV) - NLAST]:
                    tail_ev(e)
                for slot in range(2):
                    y_win(slot).wait_send()
                    y_wout(slot).wait_send()
                    x_win(slot).wait_send()
                    x_wout(slot).wait_send()
                rcopy(rows(xsend, FILL), rows(yrecv, FILL), ss.at[S_F], yr.at[0], ynb).wait_send()
                rcopy(rows(ysend, Z), rows(xrecv, Z), ss.at[S_RX], xr.at[0], xnb).wait_send()

        @pl.when(mx == 0)
        def _():
            with scope("s0_fin"):
                y_win(0).wait_send()
                y_wout(0).wait_send()
                rcopy(ysend, yrecv, ss.at[S_Y], yr.at[0], ynb).wait_send()
                pltpu.make_async_copy(big, out.at[0], ss.at[S_Z]).wait()
                rcopy(xsend, xrecv, ss.at[S_X], xr.at[0], xnb).wait_send()
                rcopy(rows(xrecv, Z), rows(xrecv, Z), ss.at[S_RY], yr.at[0], ynb).wait_send()
                rcopy(rows(xrecv, Z), rows(yrecv, Z), ss.at[S_RX], xr.at[0], xnb).wait_send()

        @pl.when(mx == 1)
        def _():
            with scope("s1_fin"):
                rcopy(rows(ysend, NDROWS), rows(yrecv, NDROWS), ss.at[S_Y], yr.at[0], ynb).wait_send()
                for e in EV[len(EV) - NLAST:]:
                    tail_ev(e)

    def fn(x_padded, Win, Wout):
        return pl.pallas_call(
            body,
            out_shape=jax.ShapeDtypeStruct((1, NB, DM), F32),
            in_specs=[pl.BlockSpec(memory_space=pl.ANY)] * 3,
            out_specs=pl.BlockSpec(memory_space=pltpu.VMEM),
            scratch_shapes=[
                pltpu.VMEM((NB, DM), F32),
                pltpu.VMEM((HALF, DM), F32),
                pltpu.VMEM((512, DM), F32),
                pltpu.VMEM((2, DM, HH), F32),
                pltpu.VMEM((2, HH, DM), F32),
                pltpu.VMEM((3, DM, 2 * HH), BF),
                pltpu.VMEM((3, 2 * HH, DM), BF),
                pltpu.VMEM((HALF, DM), BF),
                pltpu.VMEM((HALF, DM), BF),
                pltpu.VMEM((HALF, DM), BF),
                pltpu.VMEM((HALF, DM), BF),
                pltpu.VMEM((P1R, HH), BF),
            ],
            compiler_params=pltpu.CompilerParams(
                collective_id=0, vmem_limit_bytes=48 * 1024 * 1024),
        )(x_padded, Win, Wout)

    return fn


_KERNEL_CFG = {}


def pallas_dist_pipemlp_pp2tp2_xy_b4096_d256_h512_kernel(x_padded, Win, Wout):
    return make(**_KERNEL_CFG)(x_padded, Win, Wout)
```

```python
import contextlib
import jax
import jax.numpy as jnp
from jax import lax
from jax.experimental import pallas as pl
from jax.experimental.pallas import tpu as pltpu

BF = jnp.bfloat16
F32 = jnp.float32
MESH = pl.DeviceIdType.MESH

NB = 4096
DM = 256
HH = 512
HALF = 2048
CH = 64
PG = 32
NPG = HALF // PG
LN = 128


def _mlp(a, win, wout):
    h = jnp.dot(a, win, preferred_element_type=F32)
    h = jnp.maximum(h, 0.0).astype(BF)
    return jnp.dot(h, wout, preferred_element_type=F32)


def _relu_mm(a, w):
    return jnp.maximum(jnp.dot(a, w, preferred_element_type=F32), 0.0).astype(BF)


def _split(total, sizes, base=0):
    out, s, i = [], 0, 0
    while s < total:
        z = min(sizes[min(i, len(sizes) - 1)], total - s)
        out.append((base + s, z))
        s += z
        i += 1
    return out


DEFAULT = dict(
    na=2,
    nl=4,
    ua=2,
    lead=4,
    rel=(((8, 128), (9, 128), (10, 96), (11, 64)),
         ((8, 128), (9, 128), (10, 96), (12, 32), (11, 64))),
    relp=(32, 48),
    a3=(12, 13),
    ev0=("i8", "i9", "x0", "i10", "x1", "x2", "i11"),
    ev1={27: ("i8",), 29: ("i9",), 31: ("i10", "x0", "i12", "i11")},
    last_split=(64, 32, 32),
    conv_at=({9: (0, 1), 12: (2,), 13: (3,), 14: (4,), 15: (7, 8, 9)},
             {10: (0, 1), 12: (2,), 13: (3,), 15: (4,)}),
    ord1=(1, 0),
    ord0=(0, 1),
    scopes=False,
)


def make(**kw):
    cfg = dict(DEFAULT)
    cfg.update(kw)
    N1 = 6
    G0 = 8
    P1R = N1 * 128
    NLB = cfg["nl"]
    NLR = NLB * 128
    UA = cfg["ua"]
    A3 = cfg["a3"]
    LEAD = cfg["lead"]
    NE1 = cfg.get('ne1', 7)
    NS1 = cfg.get('ns1', 5)
    LL = (8 - NE1) * 256 // G0
    RELP = ([], [])
    GRP = ({}, {})
    DIR = ({}, {})
    BMSG = ({}, {})
    Z = [0, 0]
    for s in range(2):
        for (b, n) in cfg["rel"][s]:
            idx = []
            for (a, m) in _split(n, (cfg["relp"][s],)):
                idx.append(len(RELP[s]))
                RELP[s].append((Z[s] + a, m, b * 128 + a, b))
            GRP[s][b] = (Z[s], n, b * 128, idx)
            Z[s] += n
        DIR[s][0] = (0, NLR, 0, LN)
        DIR[s][1] = (0, NLR, LN, LN)
        DIR[s][2] = (NLR, P1R - NLR, 0, DM)
        for b in range(N1, 16):
            skip = GRP[s][b][1] if b in GRP[s] else 0
            if skip == 128:
                parts = []
            elif b == 15:
                parts = _split(128 - skip, cfg["last_split"], b * 128 + skip)
            else:
                parts = [(b * 128 + skip, 128 - skip)]
            BMSG[s][b] = [3 + b - N1 + t for t in range(len(parts))]
            for key, (r, n) in zip(BMSG[s][b], parts):
                DIR[s][key] = (r, n, 0, DM)
    NREL = max(len(RELP[0]), len(RELP[1]))
    A3M = {}
    for b in A3:
        assert b not in GRP[0] and G0 <= b < 15
        A3M[BMSG[0][b][0]] = b

    KL = BMSG[0][15][-1]
    BL = cfg["rel"][0][-1][0]
    assert cfg["rel"][0][-1] == cfg["rel"][1][-1] and BMSG[0][15] == BMSG[1][15]
    LAST = [f"d{KL - 1}", f"r{BL}", f"d{KL}"]

    WINP = _split(DM, cfg.get("win_pieces", (16, 48, 32, 64, 96)))
    NPA = cfg.get("npa", 3)

    def scope(name):
        if cfg["scopes"]:
            return jax.named_scope(name)
        return contextlib.nullcontext()

    def body(x_hbm, win_hbm, wout_hbm, out,
             big, pown, wfin, wfout, wbin, wbout,
             ysend, yrecv, xsend, xrecv, hbuf):
        def scoped(ld, wr, yr, xr, ss):
            inner(x_hbm, win_hbm, wout_hbm, out, big, pown, wfin, wfout, wbin, wbout,
                  ysend, yrecv, xsend, xrecv, hbuf, ld, wr, yr, xr, ss)
        pl.run_scoped(
            scoped,
            pltpu.SemaphoreType.DMA((32,)),
            pltpu.SemaphoreType.DMA((16,)),
            pltpu.SemaphoreType.DMA((NPG + NREL,)),
            pltpu.SemaphoreType.DMA((24,)),
            pltpu.SemaphoreType.DMA((16,)),
        )

    def inner(x_hbm, win_hbm, wout_hbm, out,
              big, pown, wfin, wfout, wbin, wbout,
              ysend, yrecv, xsend, xrecv, hbuf,
              ld, wr, yr, xr, ss):
        mx = lax.axis_index("x")
        my = lax.axis_index("y")
        ynb = (mx, 1 - my)
        xnb = (1 - mx, my)
        own0 = my * HALF
        oth0 = (1 - my) * HALF
        first = mx + my == 0
        bar = pltpu.get_barrier_semaphore()

        def rcopy(src, dst, ssem, rsem, dev):
            return pltpu.make_async_remote_copy(
                src_ref=src, dst_ref=dst, send_sem=ssem, recv_sem=rsem,
                device_id=dev, device_id_type=MESH)

        hb = [1 - mx, mx]
        NP = len(WINP)
        NPRO = NP - 1
        L_WO0, L_WI1, L_WO1, L_X = NP, NP + 1, NP + 2, NP + 3

        def ld_win(slot, r0, n, k):
            return pltpu.make_async_copy(
                win_hbm.at[hb[slot], pl.ds(r0, n), :], wfin.at[slot, pl.ds(r0, n), :], ld.at[k])

        def ld_wout(slot, k):
            return pltpu.make_async_copy(wout_hbm.at[hb[slot]], wfout.at[slot], ld.at[k])

        def cv_win(slot, r0, n):
            wbin[slot, pl.ds(r0, n), pl.ds(0, HH)] = wfin[slot, pl.ds(r0, n), :].astype(BF)

        def cv_wout(slot):
            wbout[slot, pl.ds(0, HH), :] = wfout[slot].astype(BF)

        def y_win(slot, r0=0, n=DM):
            return rcopy(wbin.at[slot, pl.ds(r0, n), pl.ds(0, HH)],
                         wbin.at[slot, pl.ds(r0, n), pl.ds(HH, HH)],
                         ss.at[2 * slot], wr.at[2 * slot], ynb)

        def y_wout(slot):
            return rcopy(wbout.at[slot, pl.ds(0, HH), :], wbout.at[slot, pl.ds(HH, HH), :],
                         ss.at[2 * slot + 1], wr.at[2 * slot + 1], ynb)

        def y_wout_col(c):
            return rcopy(wbout.at[1, pl.ds(0, HH), pl.ds(c * LN, LN)],
                         wbout.at[1, pl.ds(HH, HH), pl.ds(c * LN, LN)],
                         ss.at[3], wr.at[8 + c], ynb)

        def x_win(half, r0=0, n=DM):
            return rcopy(wbin.at[0, pl.ds(r0, n), pl.ds(half * HH, HH)],
                         wbin.at[2, pl.ds(r0, n), pl.ds(half * HH, HH)],
                         ss.at[4 + 2 * half], wr.at[4 + 2 * half], xnb)

        def x_wout(half):
            return rcopy(wbout.at[0, pl.ds(half * HH, HH), :], wbout.at[2, pl.ds(half * HH, HH), :],
                         ss.at[5 + 2 * half], wr.at[5 + 2 * half], xnb)

        S_Y, S_X, S_RY, S_RX = 8, 9, 10, 11
        RB = 1024

        def xload(i):
            base = oth0 if i % 2 == 0 else own0
            off = pl.multiple_of(base + (i // 2) * 256, 256)
            return pltpu.make_async_copy(
                x_hbm.at[0, pl.ds(off, 256), :], big.at[pl.ds(i * 256, 256), :], ld.at[L_X + i // 2])

        def rows(ref, n):
            return ref.at[pl.ds(0, n), :]

        def oth(r, n):
            return (0, pl.ds(pl.multiple_of(oth0 + r, 16), n), slice(None))

        def dcopy(s, j):
            r, n, c, nc = DIR[s][j]
            return rcopy(ysend.at[pl.ds(r, n), pl.ds(c, nc)], yrecv.at[pl.ds(r, n), pl.ds(c, nc)],
                         ss.at[S_Y], yr.at[j], ynb)

        def acopy(j):
            r, n, _, _ = DIR[0][j]
            return rcopy(xsend.at[pl.ds(r, n), :], xsend.at[pl.ds(r, n), :],
                         ss.at[S_Y], yr.at[j], ynb)

        def rel_in(s, b):
            a, n, o, _ = GRP[s][b]
            return rcopy(ysend.at[pl.ds(o, n), :], xrecv.at[pl.ds(a, n), :],
                         ss.at[S_RX], xr.at[b], xnb)

        def rel_y(s, j):
            a, n, _, _ = RELP[s][j]
            return rcopy(xrecv.at[pl.ds(a, n), :], xrecv.at[pl.ds(RB + a, n), :],
                         ss.at[S_RY], yr.at[NPG + j], ynb)

        def rel_x(s, j):
            a, n, o, b = RELP[s][j]
            return rcopy(xrecv.at[pl.ds(RB + a, n), :], yrecv.at[pl.ds(o, n), :],
                         ss.at[S_RX], xr.at[8 + b], xnb)

        def rel_xg(s, b):
            a, n, o, _ = GRP[s][b]
            return rcopy(xrecv.at[pl.ds(RB + a, n), :], yrecv.at[pl.ds(o, n), :],
                         ss.at[S_RX], xr.at[8 + b], xnb)

        def conv(r, n):
            out[oth(r, n)] = yrecv[pl.ds(r, n), :].astype(F32)

        def conv_msg(s, j):
            if j == 0:
                return
            conv(DIR[s][j][0], DIR[s][j][1])

        def tail_ev(s, e):
            j = int(e[1:])
            with scope("s1_e" + e):
                if e[0] == "d":
                    dcopy(s, j).wait_recv()
                    conv_msg(s, j)
                else:
                    rel_xg(s, j).wait_recv()
                    conv(GRP[s][j][2], GRP[s][j][1])

        def loads0(npre, lo=0, hi=99):
            def w(j):
                return lambda: ld_win(0, *WINP[j], j)

            def xl(i):
                return lambda: xload(i)
            seq = [w(j) for j in range(1, npre)]
            seq += [lambda: ld_win(1, 0, DM, L_WI1), xl(0), xl(1), lambda: ld_wout(1, L_WO1)]
            if npre == NPRO:
                seq += [w(NPRO), xl(2), xl(3), lambda: ld_wout(0, L_WO0)]
                seq += [xl(i) for i in range(4, 16)]
            else:
                seq += [w(j) for j in range(npre, NPRO)]
                seq += [xl(2), xl(3), w(NPRO), xl(4), xl(5)]
                seq += [lambda: ld_wout(0, L_WO0)]
                seq += [xl(i) for i in range(6, 16)]
            for c in seq[lo:hi]:
                c().start()

        ST1, ST2 = cfg.get("stag", (5, 99))

        with scope("s0_pro"):
            ld_win(0, *WINP[0], 0).start()
            pl.semaphore_signal(bar, inc=1, device_id=ynb, device_id_type=MESH)

            @pl.when(mx == 0)
            def _():
                pl.semaphore_signal(bar, inc=1, device_id=xnb, device_id_type=MESH)

                @pl.when(my == 1)
                def _():
                    loads0(NPRO)

                @pl.when(my == 0)
                def _():
                    loads0(NPA, 0, ST1)

            @pl.when(mx == 1)
            def _():
                for j in range(1, NP):
                    ld_win(0, *WINP[j], j).start()
                ld_wout(0, L_WO0).start()
                ld_win(1, 0, DM, L_WI1).start()
                ld_wout(1, L_WO1).start()
        with scope("s0_pa"):
            ld_win(0, *WINP[0], 0).wait()
            cv_win(0, *WINP[0])

            @pl.when(first)
            def _():
                for j in range(1, NPA):
                    ld_win(0, *WINP[j], j).wait()
                cv_win(0, WINP[1][0], WINP[NPA][0] - WINP[1][0])
                ld_win(1, 0, DM, L_WI1).wait()
                loads0(NPA, ST1, ST2)
                cv_win(1, 0, DM)
        with scope("s0_pb"):
            pl.semaphore_wait(bar, 1 + mx)
            y_win(0, *WINP[0]).start()
        with scope("s0_pc"):
            @pl.when(first)
            def _():
                y_win(0, WINP[1][0], WINP[NPA][0] - WINP[1][0]).start()
                loads0(NPA, ST2)

            @pl.when(jnp.logical_not(first))
            def _():
                for j in range(1, NPRO):
                    ld_win(0, *WINP[j], j).wait()
                    cv_win(0, *WINP[j])
                    y_win(0, *WINP[j]).start()

        @pl.when(mx == 0)
        def _stage0():
            W0I = (1, slice(None), pl.ds(0, HH))
            W0O = (1, pl.ds(0, HH), slice(None))

            def xwait(i):
                r = i * 512 if isinstance(i, int) else pl.multiple_of(i * 512, 512)
                pltpu.make_async_copy(
                    big.at[pl.ds(r, 512), :], big.at[pl.ds(r, 512), :], ld.at[L_X + i]).wait()

            def psend(k, n=PG):
                r = k * PG if isinstance(k, int) else pl.multiple_of(k * PG, PG)
                return rcopy(ysend.at[pl.ds(r, n), :], yrecv.at[pl.ds(r, n), :],
                             ss.at[S_Y], yr.at[k], ynb)

            def pwait(r, n):
                rcopy(ysend.at[pl.ds(r, n), :], yrecv.at[pl.ds(r, n), :],
                      ss.at[S_Y], yr.at[r // PG], ynb).wait_recv()

            def psends(i):
                for q in range(8):
                    psend(i * 8 + q).start()

            def l0_out(p, r, q):
                ysend[pl.ds(q, 256), :] = p[:256].astype(BF)
                pown[pl.ds(q, 256), :] = p[256:]

            with scope("s0_init"):
                @pl.when(my == 1)
                def _():
                    ld_win(1, 0, DM, L_WI1).wait()
                    cv_win(1, 0, DM)
                xwait(0)
            with scope("s0_h0"):
                hbuf[pl.ds(0, 512), :] = _relu_mm(big[pl.ds(0, 512), :].astype(BF), wbin[W0I])

                @pl.when(my == 1)
                def _():
                    ld_win(0, *WINP[NPRO], NPRO).wait()
                    cv_win(0, *WINP[NPRO])
                    y_win(0, *WINP[NPRO]).start()
                ld_wout(1, L_WO1).wait()
            with scope("s0_o0"):
                cv_wout(1)
                l0_out(jnp.dot(hbuf[pl.ds(0, 512), :], wbout[W0O], preferred_element_type=F32), 0, 0)

                @pl.when(my == 0)
                def _():
                    for j in range(NPA, NPRO):
                        ld_win(0, *WINP[j], j).wait()
                    cv_win(0, WINP[NPA][0], WINP[NPRO][0] - WINP[NPA][0])
                    y_win(0, WINP[NPA][0], WINP[NPRO][0] - WINP[NPA][0]).start()

            with scope("s0_l0"):
                def it(i, c):
                    r = pl.multiple_of(i * 512, 512)
                    with scope("s0_lb"):
                        xwait(i)
                        p = _mlp(big[pl.ds(r, 512), :].astype(BF), wbin[W0I], wbout[W0O])
                        l0_out(p, r, pl.multiple_of(i * 256, 256))
                    return c

                def ps(i, c):
                    psends(i)
                    return c

                def seg(sg, lo):
                    @pl.when(sg + 2 * my == 1)
                    def _():
                        with scope("s0_lp"):
                            ld_win(0, *WINP[NPRO], NPRO).wait()
                            cv_win(0, *WINP[NPRO])
                            y_win(0, *WINP[NPRO]).start()

                    @pl.when(sg + my == 2)
                    def _():
                        with scope("s0_lw"):
                            ld_wout(0, L_WO0).wait()
                            cv_wout(0)
                            y_wout(0).start()

                    @pl.when(sg + 3 * my == 2)
                    def _():
                        for k in range(LEAD):
                            psend(2 * k, CH).start()

                    @pl.when(sg + my == 3)
                    def _():
                        with scope("s0_ls"):
                            lax.fori_loop(0, NS1, ps, 0)
                    hi = jnp.where(sg == 0, 2, jnp.where(sg == 1, 3 + (NS1 - 3) * my, 8 - (8 - NE1) * my))
                    lax.fori_loop(lo, hi, it, 0)
                    return hi
                lax.fori_loop(0, 3, seg, 1)

            with scope("s0_wait_w1"):
                y_win(0).wait_recv()
                y_wout(0).wait_recv()
                x_win(0).wait_recv()

            def w2wait():
                x_wout(0).wait_recv()
                x_win(1).wait_recv()
                x_wout(1).wait_recv()

            def chunk(r, n, g3=False):
                with scope("s0_wp"):
                    pwait(r, n)
                a = (pown[pl.ds(r, n), :] + yrecv[pl.ds(r, n), :].astype(F32)).astype(BF)
                a = _mlp(a, wbin[0], wbout[0]).astype(BF)
                if g3:
                    a = _mlp(a, wbin[2], wbout[2]).astype(BF)
                xsend[pl.ds(r, n), :] = a
                rcopy(xsend.at[pl.ds(r, n), :], xrecv.at[pl.ds(r, n), :],
                      ss.at[S_X], xr.at[r // 128], xnb).start()

            def relay_ev(side, ev):
                with scope("s0_" + ev):
                    j = int(ev[1:])
                    if ev[0] == "i":
                        rel_in(side, j).wait_recv()
                        for t in GRP[side][j][3]:
                            rel_y(side, t).start()
                    else:
                        rel_y(1 - side, j).wait_recv()
                        rel_x(1 - side, j).start()
                        if 1 <= j <= 8:
                            out[0, pl.ds((j - 1) * 512, 512), :] = jnp.zeros((512, DM), F32)

            def rest_ev(side, evs):
                evs = list(evs)
                rest = [f"x{j}" for j in range(len(RELP[1 - side])) if f"x{j}" not in evs]
                assert [e for e in evs if e[0] == "i"] == [f"i{b}" for b in GRP[side]]
                assert len(RELP[1 - side]) >= 9
                return rest

            def fin0(side):
                with scope("s0_fin"):
                    y_win(0).wait_send()
                    y_wout(0).wait_send()
                    rcopy(ysend, yrecv, ss.at[S_Y], yr.at[0], ynb).wait_send()
                    rcopy(xsend, xrecv, ss.at[S_X], xr.at[0], xnb).wait_send()
                    zy, zx = Z[side], Z[1 - side]
                    rcopy(rows(xrecv, zy), rows(xrecv, zy), ss.at[S_RY], yr.at[0], ynb).wait_send()
                    if not cfg.get("fin_out", True):
                        rcopy(rows(xrecv, zx), rows(yrecv, zx), ss.at[S_RX], xr.at[0], xnb).wait_send()

            def side0():
                NIT = HALF // (PG * UA)

                def ita(j, c):
                    for u in range(UA):
                        chunk(pl.multiple_of((j * UA + u) * PG, PG), PG)

                    @pl.when(j < NIT - 2 * LEAD // UA)
                    def _():
                        for u in range(UA // 2):
                            psend(j * UA + 2 * u + 2 * LEAD, CH).start()
                    return c
                with scope("s0_p2"):
                    lax.fori_loop(0, NIT, ita, 0)
                for ev in list(cfg["ev0"]) + rest_ev(0, cfg["ev0"]):
                    relay_ev(0, ev)
                    if ev == "x0":
                        w2wait()
                fin0(0)

            def side1():
                evs = cfg["ev1"]
                rest = rest_ev(1, [e for k in sorted(evs) for e in evs[k]])
                for i in range(NS1, NE1):
                    psends(i)
                for i in range(NE1, 8):
                    xwait(i)

                def pair_late(j, c):
                    q = pl.multiple_of(NE1 * 256 + j * LL, LL)
                    rb = pl.multiple_of((q // 256) * 512 + q % 256, LL)
                    chunk(pl.multiple_of(2 * j * CH, CH), CH)
                    chunk(pl.multiple_of((2 * j + 1) * CH, CH), CH)
                    a = jnp.concatenate(
                        [big[pl.ds(rb, LL), :], big[pl.ds(pl.multiple_of(rb + 256, LL), LL), :]],
                        axis=0).astype(BF)
                    p = _mlp(a, wbin[W0I], wbout[W0O])
                    ysend[pl.ds(q, LL), :] = p[:LL].astype(BF)
                    pown[pl.ds(q, LL), :] = p[LL:]
                    for t in range(LL // PG):
                        psend(q // PG + t).start()
                    return c

                def events(j, par):
                    for k in sorted(evs):
                        if k % 2 == par and k < 31:
                            @pl.when(j == k // 2)
                            def _():
                                for ev in evs[k]:
                                    relay_ev(1, ev)

                def pair_g3(j, c):
                    chunk(pl.multiple_of(2 * j * CH, CH), CH)

                    @pl.when(j == G0)
                    def _():
                        with scope("s0_wait_w2"):
                            w2wait()
                    events(j, 0)
                    chunk(pl.multiple_of((2 * j + 1) * CH, CH), CH, True)
                    events(j, 1)
                    return c
                with scope("s0_p2a"):
                    lax.fori_loop(0, G0, pair_late, 0)
                with scope("s0_p2b"):
                    lax.fori_loop(G0, 16, pair_g3, 0)
                for ev in list(evs[31]) + rest:
                    relay_ev(1, ev)
                fin0(1)

            for side in cfg["ord0"]:
                pl.when(my == side)((side0, side1)[side])

        @pl.when(mx == 1)
        def _stage1():
            a3 = xsend
            with scope("s1_init"):
                x_win(0, 0, WINP[NPRO][0]).start()
                ld_win(0, *WINP[NPRO], NPRO).wait()
                cv_win(0, *WINP[NPRO])
                y_win(0, *WINP[NPRO]).start()
                x_win(0, *WINP[NPRO]).start()
                ld_wout(0, L_WO0).wait()
                cv_wout(0)
                y_wout(0).start()
                x_wout(0).start()
                ld_win(1, 0, DM, L_WI1).wait()
                cv_win(1, 0, DM)
                y_win(1).start()
                ld_wout(1, L_WO1).wait()
                cv_wout(1)
                y_wout_col(0).start()
                y_wout_col(1).start()
            with scope("s1_wait_w2"):
                y_win(0).wait_recv()
                x_win(1).start()
                y_wout(0).wait_recv()
                x_wout(1).start()

            def wait_a2(b):
                r = b * 128 if isinstance(b, int) else pl.multiple_of(b * 128, 128)
                with scope("s1_wa"):
                    rcopy(xsend.at[pl.ds(r, 128), :], xrecv.at[pl.ds(r, 128), :],
                          ss.at[S_X], xr.at[b], xnb).wait_recv()

            def own(r, n, c=0, nc=DM):
                return (0, pl.ds(pl.multiple_of(own0 + r, 16), n), pl.ds(c, nc))

            W3I_L = (1, slice(None), pl.ds(0, HH))
            W3I_R = (1, slice(None), pl.ds(HH, HH))
            W3O_L = (1, pl.ds(0, HH), slice(None))

            def p1(i, c):
                wait_a2(i)
                r = pl.multiple_of(i * 128, 128)
                v = _mlp(xrecv[pl.ds(r, 128), :], wbin[0], wbout[0]).astype(BF)
                a3[pl.ds(r, 128), :] = v
                pown[pl.ds(r, 128), :] = _mlp(v, wbin[W3I_L], wbout[W3O_L])
                return c

            def orem(j):
                r, n, c, nc = DIR[0][j]
                o = pown[pl.ds(r, n), pl.ds(c, nc)] + jnp.dot(
                    hbuf[pl.ds(r, n), :], wbout[1, pl.ds(HH, HH), pl.ds(c, nc)],
                    preferred_element_type=F32)
                out[own(r, n, c, nc)] = o
                ysend[pl.ds(r, n), pl.ds(c, nc)] = o.astype(BF)
                dcopy(0, j).start()

            def p1h(i, c):
                wait_a2(i)
                r = pl.multiple_of(i * 128, 128)
                v = _mlp(xrecv[pl.ds(r, 128), :], wbin[0], wbout[0]).astype(BF)
                h = _relu_mm(v, wbin[1])
                hbuf[pl.ds(r, 128), :] = h[:, HH:]
                pown[pl.ds(r, 128), :] = jnp.dot(h[:, :HH], wbout[W3O_L], preferred_element_type=F32)

                @pl.when(i == NLB - 1)
                def _():
                    with scope("s1_ol"):
                        y_wout_col(0).wait_recv()
                        orem(0)
                return c

            NA = cfg["na"]
            def p12():
                with scope("s1_p1a"):
                    lax.fori_loop(0, NA, p1, 0)
                with scope("s1_wait_w3i"):
                    y_win(1).wait_recv()
                with scope("s1_hr"):
                    hbuf[pl.ds(0, NA * 128), :] = _relu_mm(a3[pl.ds(0, NA * 128), :], wbin[W3I_R])
                with scope("s1_p1b"):
                    lax.fori_loop(NA, N1, p1h, 0)
                with scope("s1_wait_w3"):
                    y_wout_col(1).wait_recv()
                with scope("s1_p2"):
                    orem(1)
                    orem(2)
                for b in range(N1, G0):
                    with scope(f"s1_b{b}"):
                        blk(b, None)

            def blk(b, side, msgs=()):
                r = b * 128
                s = 0 if side is None else side
                wait_a2(b)
                for j in msgs:
                    dcopy(1 - s, j).wait_recv()
                if side == 1:
                    v = _mlp(xrecv[pl.ds(r, CH), :], wbin[0], wbout[0]).astype(BF)
                    v = jnp.concatenate([v, xrecv[pl.ds(r + CH, CH), :]], axis=0)
                else:
                    v = _mlp(xrecv[pl.ds(r, 128), :], wbin[0], wbout[0]).astype(BF)
                if side == 0 and b in A3:
                    a3[pl.ds(r, 128), :] = v
                else:
                    o = _mlp(v, wbin[1], wbout[1])
                    out[own(r, 128)] = o
                    ysend[pl.ds(r, 128), :] = o.astype(BF)
                for j in msgs:
                    conv_msg(1 - s, j)
                if side == 0 and b in A3:
                    acopy(BMSG[0][b][0]).start()
                else:
                    if b in GRP[s]:
                        rel_in(s, b).start()
                    for j in BMSG[s][b]:
                        dcopy(s, j).start()

            DUP = cfg.get("dup", True)
            if not DUP:
                p12()

            def p3(side):
                if DUP:
                    p12()
                for b in range(G0, 16):
                    with scope(f"s1_b{b}"):
                        blk(b, side, cfg["conv_at"][side].get(b, ()))
                if side == 1:
                    for j in A3M:
                        acopy(j).wait_recv()

            for side in cfg["ord1"]:
                pl.when(my == side)(lambda side=side: p3(side))
            with scope("s1_l3"):
                for b in A3:
                    out[0, pl.ds(b * 128, 128), :] = _mlp(a3[pl.ds(b * 128, 128), :], wbin[1], wbout[1])

            def tail(side):
                s = 1 - side
                done = [j for v in cfg["conv_at"][side].values() for j in v]
                assert len(set(done)) == len(done) and all(j in DIR[s] for j in done)
                assert not (side == 1 and any(j in A3M for j in done))
                ev = []
                rem = 0
                for j in reversed(list(DIR[s])):
                    if j not in done and not (side == 1 and j in A3M):
                        ev.append((-rem, f"d{j}"))
                    rem += DIR[s][j][1]
                rem = cfg.get("relay_early", (32, 0))[side]
                for b in reversed(list(GRP[s])):
                    ev.append((-rem, f"r{b}"))
                    rem += GRP[s][b][1]
                ev.sort()
                for _, e in ev:
                    if e not in LAST:
                        tail_ev(s, e)
                z = Z[side]
                rcopy(rows(ysend, z), rows(xrecv, z), ss.at[S_RX], xr.at[0], xnb).wait_send()

            with scope("s1_tail"):
                for slot in range(2):
                    y_win(slot).wait_send()
                    y_wout(slot).wait_send()
                    x_win(slot).wait_send()
                    x_wout(slot).wait_send()
                for side in cfg.get("ordt", (1, 0)):
                    pl.when(my == side)(lambda side=side: tail(side))

        if cfg.get("fin_out", True):
            for side in range(2):
                @pl.when(mx + 2 * my == 2 * side)
                def _():
                    zx = Z[1 - side]
                    rcopy(rows(xrecv, zx), rows(yrecv, zx), ss.at[S_RX], xr.at[0], xnb).wait_send()

        @pl.when(mx == 1)
        def _():
            with scope("s1_fin"):
                for e in LAST[:-1]:
                    tail_ev(0, e)
                for side in range(2):
                    @pl.when(my == side)
                    def _():
                        n = HALF - Z[side]
                        rcopy(rows(ysend, n), rows(yrecv, n), ss.at[S_Y], yr.at[0], ynb).wait_send()
                tail_ev(0, LAST[-1])

    def fn(x_padded, Win, Wout):
        return pl.pallas_call(
            body,
            out_shape=jax.ShapeDtypeStruct((1, NB, DM), F32),
            in_specs=[pl.BlockSpec(memory_space=pl.ANY)] * 3,
            out_specs=pl.BlockSpec(memory_space=pltpu.VMEM),
            scratch_shapes=[
                pltpu.VMEM((NB, DM), F32),
                pltpu.VMEM((HALF, DM), F32),
                pltpu.VMEM((2, DM, HH), F32),
                pltpu.VMEM((2, HH, DM), F32),
                pltpu.VMEM((3, DM, 2 * HH), BF),
                pltpu.VMEM((3, 2 * HH, DM), BF),
                pltpu.VMEM((HALF, DM), BF),
                pltpu.VMEM((HALF, DM), BF),
                pltpu.VMEM((HALF, DM), BF),
                pltpu.VMEM((HALF, DM), BF),
                pltpu.VMEM((P1R, HH), BF),
            ],
            compiler_params=pltpu.CompilerParams(
                collective_id=0, vmem_limit_bytes=48 * 1024 * 1024),
        )(x_padded, Win, Wout)

    return fn


_KERNEL_CFG = {}


def pallas_dist_pipemlp_pp2tp2_xy_b4096_d256_h512_kernel(x_padded, Win, Wout):
    return make(**_KERNEL_CFG)(x_padded, Win, Wout)
```

```python
import contextlib
import jax
import jax.numpy as jnp
from jax import lax
from jax.experimental import pallas as pl
from jax.experimental.pallas import tpu as pltpu

BF = jnp.bfloat16
F32 = jnp.float32
MESH = pl.DeviceIdType.MESH

NB = 4096
DM = 256
HH = 512
HALF = 2048
CH = 64
PG = 32
NPG = HALF // PG
LN = 128


def _mlp(a, win, wout):
    h = jnp.dot(a, win, preferred_element_type=F32)
    h = jnp.maximum(h, 0.0).astype(BF)
    return jnp.dot(h, wout, preferred_element_type=F32)


def _relu_mm(a, w):
    return jnp.maximum(jnp.dot(a, w, preferred_element_type=F32), 0.0).astype(BF)


def _split(total, sizes, base=0):
    out, s, i = [], 0, 0
    while s < total:
        z = min(sizes[min(i, len(sizes) - 1)], total - s)
        out.append((base + s, z))
        s += z
        i += 1
    return out


DEFAULT = dict(
    na=2,
    nl=4,
    ua=2,
    lead=4,
    rel=(((8, 128), (9, 128), (10, 96), (11, 64)),
         ((8, 128), (9, 128), (10, 96), (12, 32), (11, 64))),
    relp=(32, 48),
    a3=(12, 13),
    ev0=("i8", "i9", "x0", "i10", "x1", "x2", "i11"),
    ev1={27: ("i8",), 29: ("i9",), 31: ("i10", "x0", "i12", "i11")},
    last_split=(64, 32, 32),
    conv_at=({9: (0, 1), 12: (2,), 13: (3,), 14: (4,), 15: (7, 8, 9)},
             {10: (0, 1), 12: (2,), 13: (3,), 15: (4,)}),
    ord1=(1, 0),
    ord0=(0, 1),
    scopes=False,
)


def make(**kw):
    cfg = dict(DEFAULT)
    cfg.update(kw)
    N1 = 6
    G0 = 8
    P1R = N1 * 128
    NLB = cfg["nl"]
    NLR = NLB * 128
    UA = cfg["ua"]
    A3 = cfg["a3"]
    LEAD = cfg["lead"]
    NE1 = cfg.get('ne1', 7)
    NS1 = cfg.get('ns1', 5)
    LL = (8 - NE1) * 256 // G0
    RELP = ([], [])
    GRP = ({}, {})
    DIR = ({}, {})
    BMSG = ({}, {})
    Z = [0, 0]
    for s in range(2):
        for (b, n) in cfg["rel"][s]:
            idx = []
            for (a, m) in _split(n, (cfg["relp"][s],)):
                idx.append(len(RELP[s]))
                RELP[s].append((Z[s] + a, m, b * 128 + a, b))
            GRP[s][b] = (Z[s], n, b * 128, idx)
            Z[s] += n
        DIR[s][0] = (0, NLR, 0, LN)
        DIR[s][1] = (0, NLR, LN, LN)
        DIR[s][2] = (NLR, P1R - NLR, 0, DM)
        for b in range(N1, 16):
            skip = GRP[s][b][1] if b in GRP[s] else 0
            if skip == 128:
                parts = []
            elif b == 15:
                parts = _split(128 - skip, cfg["last_split"], b * 128 + skip)
            else:
                parts = [(b * 128 + skip, 128 - skip)]
            BMSG[s][b] = [3 + b - N1 + t for t in range(len(parts))]
            for key, (r, n) in zip(BMSG[s][b], parts):
                DIR[s][key] = (r, n, 0, DM)
    NREL = max(len(RELP[0]), len(RELP[1]))
    A3M = {}
    for b in A3:
        assert b not in GRP[0] and G0 <= b < 15
        A3M[BMSG[0][b][0]] = b

    KL = BMSG[0][15][-1]
    BL = cfg["rel"][0][-1][0]
    assert cfg["rel"][0][-1] == cfg["rel"][1][-1] and BMSG[0][15] == BMSG[1][15]
    LAST = [f"d{KL - 1}", f"r{BL}", f"d{KL}"]

    WINP = _split(DM, cfg.get("win_pieces", (16, 48, 32, 64, 96)))
    NPA = cfg.get("npa", 3)

    def scope(name):
        if cfg["scopes"]:
            return jax.named_scope(name)
        return contextlib.nullcontext()

    def body(x_hbm, win_hbm, wout_hbm, out,
             big, pown, wfin, wfout, wbin, wbout,
             ysend, yrecv, xsend, xrecv, hbuf, wfr):
        def scoped(ld, wr, yr, xr, ss):
            inner(x_hbm, win_hbm, wout_hbm, out, big, pown, wfin, wfout, wbin, wbout,
                  ysend, yrecv, xsend, xrecv, hbuf, wfr, ld, wr, yr, xr, ss)
        pl.run_scoped(
            scoped,
            pltpu.SemaphoreType.DMA((32,)),
            pltpu.SemaphoreType.DMA((16,)),
            pltpu.SemaphoreType.DMA((NPG + NREL,)),
            pltpu.SemaphoreType.DMA((24,)),
            pltpu.SemaphoreType.DMA((16,)),
        )

    def inner(x_hbm, win_hbm, wout_hbm, out,
              big, pown, wfin, wfout, wbin, wbout,
              ysend, yrecv, xsend, xrecv, hbuf, wfr,
              ld, wr, yr, xr, ss):
        mx = lax.axis_index("x")
        my = lax.axis_index("y")
        ynb = (mx, 1 - my)
        xnb = (1 - mx, my)
        own0 = my * HALF
        oth0 = (1 - my) * HALF
        first = mx + my == 0
        bar = pltpu.get_barrier_semaphore()

        def rcopy(src, dst, ssem, rsem, dev):
            return pltpu.make_async_remote_copy(
                src_ref=src, dst_ref=dst, send_sem=ssem, recv_sem=rsem,
                device_id=dev, device_id_type=MESH)

        hb = [1 - mx, mx]
        NP = len(WINP)
        NPRO = NP - 1
        L_WO0, L_WI1, L_WO1, L_X = NP, NP + 1, NP + 2, NP + 3

        def ld_win(slot, r0, n, k):
            return pltpu.make_async_copy(
                win_hbm.at[hb[slot], pl.ds(r0, n), :], wfin.at[slot, pl.ds(r0, n), :], ld.at[k])

        def ld_wout(slot, k):
            return pltpu.make_async_copy(wout_hbm.at[hb[slot]], wfout.at[slot], ld.at[k])

        def cv_win(slot, r0, n):
            wbin[slot, pl.ds(r0, n), pl.ds(0, HH)] = wfin[slot, pl.ds(r0, n), :].astype(BF)

        def cv_wout(slot):
            wbout[slot, pl.ds(0, HH), :] = wfout[slot].astype(BF)

        def y_win(slot, r0=0, n=DM):
            return rcopy(wbin.at[slot, pl.ds(r0, n), pl.ds(0, HH)],
                         wbin.at[slot, pl.ds(r0, n), pl.ds(HH, HH)],
                         ss.at[2 * slot], wr.at[2 * slot], ynb)

        FC = cfg.get("fc", (256, 128))
        R0 = WINP[0][1]

        def y_p0(st, part):
            c, n = ((0, FC[st]), (FC[st], HH - FC[st]))[part]
            return rcopy(wbin.at[0, pl.ds(0, R0), pl.ds(c, n)], wbin.at[0, pl.ds(0, R0), pl.ds(HH + c, n)],
                         ss.at[12 + part], wr.at[10 + part], ynb)

        def y_p0f(st):
            return rcopy(win_hbm.at[hb[0], pl.ds(0, R0), pl.ds(0, FC[st])], wfr.at[:, pl.ds(0, FC[st])],
                         ss.at[12], wr.at[10], ynb)

        def p0_recv(st):
            if FC[st]:
                @pl.when(my == 0)
                def _():
                    y_p0f(st).wait_recv()
                    y_p0(st, 0).wait_send()
                    wbin[0, pl.ds(0, R0), pl.ds(HH, FC[st])] = wfr[:, pl.ds(0, FC[st])].astype(BF)

                @pl.when(my == 1)
                def _():
                    y_p0(st, 0).wait_recv()
                    y_p0f(st).wait_send()
            y_p0(st, 1).wait()

        def y_wout(slot):
            return rcopy(wbout.at[slot, pl.ds(0, HH), :], wbout.at[slot, pl.ds(HH, HH), :],
                         ss.at[2 * slot + 1], wr.at[2 * slot + 1], ynb)

        def y_wout_col(c):
            return rcopy(wbout.at[1, pl.ds(0, HH), pl.ds(c * LN, LN)],
                         wbout.at[1, pl.ds(HH, HH), pl.ds(c * LN, LN)],
                         ss.at[3], wr.at[8 + c], ynb)

        def x_win(half, r0=0, n=DM):
            return rcopy(wbin.at[0, pl.ds(r0, n), pl.ds(half * HH, HH)],
                         wbin.at[2, pl.ds(r0, n), pl.ds(half * HH, HH)],
                         ss.at[4 + 2 * half], wr.at[4 + 2 * half], xnb)

        def x_wout(half):
            return rcopy(wbout.at[0, pl.ds(half * HH, HH), :], wbout.at[2, pl.ds(half * HH, HH), :],
                         ss.at[5 + 2 * half], wr.at[5 + 2 * half], xnb)

        S_Y, S_X, S_RY, S_RX = 8, 9, 10, 11
        RB = 1024

        def xload(i):
            base = oth0 if i % 2 == 0 else own0
            off = pl.multiple_of(base + (i // 2) * 256, 256)
            return pltpu.make_async_copy(
                x_hbm.at[0, pl.ds(off, 256), :], big.at[pl.ds(i * 256, 256), :],
                ld.at[L_X + (i // 2 if i else 8)])

        def hhalf(t, c=0):
            r = t * 256 if isinstance(t, int) else pl.multiple_of(t * 256, 256)
            pltpu.make_async_copy(
                big.at[pl.ds(r, 256), :], big.at[pl.ds(r, 256), :], ld.at[L_X + 8 * (1 - t)]).wait()
            hbuf[pl.ds(r, 256), :] = _relu_mm(big[pl.ds(r, 256), :].astype(BF), wbin[1, :, pl.ds(0, HH)])
            return c

        def rows(ref, n):
            return ref.at[pl.ds(0, n), :]

        def oth(r, n):
            return (0, pl.ds(pl.multiple_of(oth0 + r, 16), n), slice(None))

        def dcopy(s, j):
            r, n, c, nc = DIR[s][j]
            return rcopy(ysend.at[pl.ds(r, n), pl.ds(c, nc)], yrecv.at[pl.ds(r, n), pl.ds(c, nc)],
                         ss.at[S_Y], yr.at[j], ynb)

        def acopy(j):
            r, n, _, _ = DIR[0][j]
            return rcopy(xsend.at[pl.ds(r, n), :], xsend.at[pl.ds(r, n), :],
                         ss.at[S_Y], yr.at[j], ynb)

        def rel_in(s, b):
            a, n, o, _ = GRP[s][b]
            return rcopy(ysend.at[pl.ds(o, n), :], xrecv.at[pl.ds(a, n), :],
                         ss.at[S_RX], xr.at[b], xnb)

        def rel_y(s, j):
            a, n, _, _ = RELP[s][j]
            return rcopy(xrecv.at[pl.ds(a, n), :], xrecv.at[pl.ds(RB + a, n), :],
                         ss.at[S_RY], yr.at[NPG + j], ynb)

        def rel_x(s, j):
            a, n, o, b = RELP[s][j]
            return rcopy(xrecv.at[pl.ds(RB + a, n), :], yrecv.at[pl.ds(o, n), :],
                         ss.at[S_RX], xr.at[8 + b], xnb)

        def rel_xg(s, b):
            a, n, o, _ = GRP[s][b]
            return rcopy(xrecv.at[pl.ds(RB + a, n), :], yrecv.at[pl.ds(o, n), :],
                         ss.at[S_RX], xr.at[8 + b], xnb)

        def conv(r, n):
            out[oth(r, n)] = yrecv[pl.ds(r, n), :].astype(F32)

        def conv_msg(s, j):
            if j == 0:
                return
            conv(DIR[s][j][0], DIR[s][j][1])

        def tail_ev(s, e):
            j = int(e[1:])
            with scope("s1_e" + e):
                if e[0] == "d":
                    dcopy(s, j).wait_recv()
                    conv_msg(s, j)
                else:
                    rel_xg(s, j).wait_recv()
                    conv(GRP[s][j][2], GRP[s][j][1])

        def loads0(npre, lo=0, hi=99):
            def w(j):
                return lambda: ld_win(0, *WINP[j], j)

            def xl(i):
                return lambda: xload(i)
            if npre == NPRO:
                seq = [w(j) for j in range(1, npre)]
                seq += [lambda: ld_win(1, 0, DM, L_WI1), xl(0), xl(1), lambda: ld_wout(1, L_WO1)]
                seq += [w(NPRO), xl(2), xl(3), lambda: ld_wout(0, L_WO0)]
                seq += [xl(i) for i in range(4, 16)]
            else:
                seq = [lambda: ld_win(1, 0, DM, L_WI1), xl(0)]
                seq += [w(j) for j in range(1, npre)]
                seq += [xl(1), lambda: ld_wout(1, L_WO1)]
                seq += [w(j) for j in range(npre, NPRO)]
                seq += [xl(2), xl(3), w(NPRO), xl(4), xl(5)]
                seq += [lambda: ld_wout(0, L_WO0)]
                seq += [xl(i) for i in range(6, 16)]
            for c in seq[lo:hi]:
                c().start()

        ST0, ST1, ST2 = cfg.get("stag", (2, 4, 6))

        with scope("s0_pro"):
            ld_win(0, *WINP[0], 0).start()
            pl.semaphore_signal(bar, inc=1, device_id=ynb, device_id_type=MESH)

            @pl.when(mx == 0)
            def _():
                pl.semaphore_signal(bar, inc=1, device_id=xnb, device_id_type=MESH)

                @pl.when(my == 1)
                def _():
                    if FC[0]:
                        pl.semaphore_wait(bar, 1)
                        y_p0f(0).start()
                    loads0(NPRO)

                @pl.when(my == 0)
                def _():
                    loads0(NPA, 0, ST0)

            @pl.when(mx == 1)
            def _():
                seq = [lambda j=j: ld_win(0, *WINP[j], j) for j in range(1, NP)]
                seq += [lambda: ld_wout(0, L_WO0), lambda: ld_win(1, 0, DM, L_WI1), lambda: ld_wout(1, L_WO1)]
                k = cfg.get("dpre", 1)
                for c in seq[:k]:
                    c().start()
                if FC[1]:
                    @pl.when(my == 1)
                    def _():
                        pl.semaphore_wait(bar, 2)
                        y_p0f(1).start()
                for c in seq[k:]:
                    c().start()
        with scope("s0_pa"):
            ld_win(0, *WINP[0], 0).wait()
            cv_win(0, *WINP[0])

            @pl.when(first)
            def _():
                loads0(NPA, ST0, ST1)
                with scope("s0_pw"):
                    ld_win(1, 0, DM, L_WI1).wait()
                loads0(NPA, ST1, ST2)
                cv_win(1, 0, DM)
                with scope("s0_ph"):
                    hhalf(0)
                for j in range(1, NPA):
                    ld_win(0, *WINP[j], j).wait()
                cv_win(0, WINP[1][0], WINP[NPA][0] - WINP[1][0])
        with scope("s0_pb"):
            for st in range(2):
                @pl.when(mx == st)
                def _():
                    if FC[st]:
                        @pl.when(my == 0)
                        def _():
                            pl.semaphore_wait(bar, 1 + st)
                            y_p0(st, 0).start()
                    else:
                        pl.semaphore_wait(bar, 1 + st)
                    y_p0(st, 1).start()
        with scope("s0_pc"):
            @pl.when(first)
            def _():
                y_win(0, WINP[1][0], WINP[NPA][0] - WINP[1][0]).start()
                loads0(NPA, ST2)

            @pl.when(jnp.logical_not(first))
            def _():
                for j in range(1, NPRO):
                    ld_win(0, *WINP[j], j).wait()
                    cv_win(0, *WINP[j])
                    y_win(0, *WINP[j]).start()

        @pl.when(mx == 0)
        def _stage0():
            W0I = (1, slice(None), pl.ds(0, HH))
            W0O = (1, pl.ds(0, HH), slice(None))

            def xwait(i):
                r = i * 512 if isinstance(i, int) else pl.multiple_of(i * 512, 512)
                pltpu.make_async_copy(
                    big.at[pl.ds(r, 512), :], big.at[pl.ds(r, 512), :], ld.at[L_X + i]).wait()

            def psend(k, n=PG):
                r = k * PG if isinstance(k, int) else pl.multiple_of(k * PG, PG)
                return rcopy(ysend.at[pl.ds(r, n), :], yrecv.at[pl.ds(r, n), :],
                             ss.at[S_Y], yr.at[k], ynb)

            def pwait(r, n):
                rcopy(ysend.at[pl.ds(r, n), :], yrecv.at[pl.ds(r, n), :],
                      ss.at[S_Y], yr.at[r // PG], ynb).wait_recv()

            def psends(i):
                for q in range(8):
                    psend(i * 8 + q).start()

            def l0_out(p, r, q):
                ysend[pl.ds(q, 256), :] = p[:256].astype(BF)
                pown[pl.ds(q, 256), :] = p[256:]

            with scope("s0_init"):
                @pl.when(my == 1)
                def _():
                    ld_win(1, 0, DM, L_WI1).wait()
                    cv_win(1, 0, DM)
            with scope("s0_h0"):
                lax.fori_loop(1 - my, 2, hhalf, 0)

                @pl.when(my == 1)
                def _():
                    ld_win(0, *WINP[NPRO], NPRO).wait()
                    cv_win(0, *WINP[NPRO])
                    y_win(0, *WINP[NPRO]).start()
                ld_wout(1, L_WO1).wait()
            with scope("s0_o0"):
                cv_wout(1)
                l0_out(jnp.dot(hbuf[pl.ds(0, 512), :], wbout[W0O], preferred_element_type=F32), 0, 0)

                @pl.when(my == 0)
                def _():
                    for j in range(NPA, NPRO):
                        ld_win(0, *WINP[j], j).wait()
                    cv_win(0, WINP[NPA][0], WINP[NPRO][0] - WINP[NPA][0])
                    y_win(0, WINP[NPA][0], WINP[NPRO][0] - WINP[NPA][0]).start()

            with scope("s0_l0"):
                def it(i, c):
                    r = pl.multiple_of(i * 512, 512)
                    with scope("s0_lb"):
                        xwait(i)
                        p = _mlp(big[pl.ds(r, 512), :].astype(BF), wbin[W0I], wbout[W0O])
                        l0_out(p, r, pl.multiple_of(i * 256, 256))
                    return c

                def ps(i, c):
                    psends(i)
                    return c

                def seg(sg, lo):
                    @pl.when(sg + 2 * my == 1)
                    def _():
                        with scope("s0_lp"):
                            ld_win(0, *WINP[NPRO], NPRO).wait()
                            cv_win(0, *WINP[NPRO])
                            y_win(0, *WINP[NPRO]).start()

                    @pl.when(sg + my == 2)
                    def _():
                        with scope("s0_lw"):
                            p0_recv(0)
                            ld_wout(0, L_WO0).wait()
                            cv_wout(0)
                            y_wout(0).start()

                    @pl.when(sg + 3 * my == 2)
                    def _():
                        for k in range(LEAD):
                            psend(2 * k, CH).start()

                    @pl.when(sg + my == 3)
                    def _():
                        with scope("s0_ls"):
                            lax.fori_loop(0, NS1, ps, 0)
                    hi = jnp.where(sg == 0, 2, jnp.where(sg == 1, 3 + (NS1 - 3) * my, 8 - (8 - NE1) * my))
                    lax.fori_loop(lo, hi, it, 0)
                    return hi
                lax.fori_loop(0, 3, seg, 1)

            with scope("s0_wait_w1"):
                y_win(0, R0, DM - R0).wait_recv()
                y_wout(0).wait_recv()
                x_win(0).wait_recv()

            def w2wait():
                x_wout(0).wait_recv()
                x_win(1).wait_recv()
                x_wout(1).wait_recv()

            def chunk(r, n, g3=False):
                with scope("s0_wp"):
                    pwait(r, n)
                a = (pown[pl.ds(r, n), :] + yrecv[pl.ds(r, n), :].astype(F32)).astype(BF)
                a = _mlp(a, wbin[0], wbout[0]).astype(BF)
                if g3:
                    a = _mlp(a, wbin[2], wbout[2]).astype(BF)
                xsend[pl.ds(r, n), :] = a
                rcopy(xsend.at[pl.ds(r, n), :], xrecv.at[pl.ds(r, n), :],
                      ss.at[S_X], xr.at[r // 128], xnb).start()

            def relay_ev(side, ev):
                with scope("s0_" + ev):
                    j = int(ev[1:])
                    if ev[0] == "i":
                        rel_in(side, j).wait_recv()
                        for t in GRP[side][j][3]:
                            rel_y(side, t).start()
                    else:
                        rel_y(1 - side, j).wait_recv()
                        rel_x(1 - side, j).start()
                        if 1 <= j <= 8:
                            out[0, pl.ds((j - 1) * 512, 512), :] = jnp.zeros((512, DM), F32)

            def rest_ev(side, evs):
                evs = list(evs)
                rest = [f"x{j}" for j in range(len(RELP[1 - side])) if f"x{j}" not in evs]
                assert [e for e in evs if e[0] == "i"] == [f"i{b}" for b in GRP[side]]
                assert len(RELP[1 - side]) >= 9
                return rest

            def fin0(side):
                with scope("s0_fin"):
                    y_win(0, R0, DM - R0).wait_send()
                    y_wout(0).wait_send()
                    rcopy(ysend, yrecv, ss.at[S_Y], yr.at[0], ynb).wait_send()
                    rcopy(xsend, xrecv, ss.at[S_X], xr.at[0], xnb).wait_send()
                    zy, zx = Z[side], Z[1 - side]
                    rcopy(rows(xrecv, zy), rows(xrecv, zy), ss.at[S_RY], yr.at[0], ynb).wait_send()
                    if not cfg.get("fin_out", True):
                        rcopy(rows(xrecv, zx), rows(yrecv, zx), ss.at[S_RX], xr.at[0], xnb).wait_send()

            def side0():
                NIT = HALF // (PG * UA)

                def ita(j, c):
                    for u in range(UA):
                        chunk(pl.multiple_of((j * UA + u) * PG, PG), PG)

                    @pl.when(j < NIT - 2 * LEAD // UA)
                    def _():
                        for u in range(UA // 2):
                            psend(j * UA + 2 * u + 2 * LEAD, CH).start()
                    return c
                with scope("s0_p2"):
                    lax.fori_loop(0, NIT, ita, 0)
                for ev in list(cfg["ev0"]) + rest_ev(0, cfg["ev0"]):
                    relay_ev(0, ev)
                    if ev == "x0":
                        w2wait()
                fin0(0)

            def side1():
                evs = cfg["ev1"]
                rest = rest_ev(1, [e for k in sorted(evs) for e in evs[k]])
                for i in range(NS1, NE1):
                    psends(i)
                for i in range(NE1, 8):
                    xwait(i)

                def pair_late(j, c):
                    q = pl.multiple_of(NE1 * 256 + j * LL, LL)
                    rb = pl.multiple_of((q // 256) * 512 + q % 256, LL)
                    chunk(pl.multiple_of(2 * j * CH, CH), CH)
                    chunk(pl.multiple_of((2 * j + 1) * CH, CH), CH)
                    a = jnp.concatenate(
                        [big[pl.ds(rb, LL), :], big[pl.ds(pl.multiple_of(rb + 256, LL), LL), :]],
                        axis=0).astype(BF)
                    p = _mlp(a, wbin[W0I], wbout[W0O])
                    ysend[pl.ds(q, LL), :] = p[:LL].astype(BF)
                    pown[pl.ds(q, LL), :] = p[LL:]
                    for t in range(LL // PG):
                        psend(q // PG + t).start()
                    return c

                def events(j, par):
                    for k in sorted(evs):
                        if k % 2 == par and k < 31:
                            @pl.when(j == k // 2)
                            def _():
                                for ev in evs[k]:
                                    relay_ev(1, ev)

                def pair_g3(j, c):
                    chunk(pl.multiple_of(2 * j * CH, CH), CH)

                    @pl.when(j == G0)
                    def _():
                        with scope("s0_wait_w2"):
                            w2wait()
                    events(j, 0)
                    chunk(pl.multiple_of((2 * j + 1) * CH, CH), CH, True)
                    events(j, 1)
                    return c
                with scope("s0_p2a"):
                    lax.fori_loop(0, G0, pair_late, 0)
                with scope("s0_p2b"):
                    lax.fori_loop(G0, 16, pair_g3, 0)
                for ev in list(evs[31]) + rest:
                    relay_ev(1, ev)
                fin0(1)

            for side in cfg["ord0"]:
                pl.when(my == side)((side0, side1)[side])

        @pl.when(mx == 1)
        def _stage1():
            a3 = xsend
            with scope("s1_init"):
                x_win(0, 0, WINP[NPRO][0]).start()
                ld_win(0, *WINP[NPRO], NPRO).wait()
                cv_win(0, *WINP[NPRO])
                y_win(0, *WINP[NPRO]).start()
                x_win(0, *WINP[NPRO]).start()
                ld_wout(0, L_WO0).wait()
                cv_wout(0)
                y_wout(0).start()
                x_wout(0).start()
                ld_win(1, 0, DM, L_WI1).wait()
                cv_win(1, 0, DM)
                y_win(1).start()
                ld_wout(1, L_WO1).wait()
                cv_wout(1)
                y_wout_col(0).start()
                y_wout_col(1).start()
            with scope("s1_wait_w2"):
                p0_recv(1)
                y_win(0, R0, DM - R0).wait_recv()
                x_win(1).start()
                y_wout(0).wait_recv()
                x_wout(1).start()

            def wait_a2(b):
                r = b * 128 if isinstance(b, int) else pl.multiple_of(b * 128, 128)
                with scope("s1_wa"):
                    rcopy(xsend.at[pl.ds(r, 128), :], xrecv.at[pl.ds(r, 128), :],
                          ss.at[S_X], xr.at[b], xnb).wait_recv()

            def own(r, n, c=0, nc=DM):
                return (0, pl.ds(pl.multiple_of(own0 + r, 16), n), pl.ds(c, nc))

            W3I_L = (1, slice(None), pl.ds(0, HH))
            W3I_R = (1, slice(None), pl.ds(HH, HH))
            W3O_L = (1, pl.ds(0, HH), slice(None))

            def p1(i, c):
                wait_a2(i)
                r = pl.multiple_of(i * 128, 128)
                v = _mlp(xrecv[pl.ds(r, 128), :], wbin[0], wbout[0]).astype(BF)
                a3[pl.ds(r, 128), :] = v
                pown[pl.ds(r, 128), :] = _mlp(v, wbin[W3I_L], wbout[W3O_L])
                return c

            def orem(j):
                r, n, c, nc = DIR[0][j]
                o = pown[pl.ds(r, n), pl.ds(c, nc)] + jnp.dot(
                    hbuf[pl.ds(r, n), :], wbout[1, pl.ds(HH, HH), pl.ds(c, nc)],
                    preferred_element_type=F32)
                out[own(r, n, c, nc)] = o
                ysend[pl.ds(r, n), pl.ds(c, nc)] = o.astype(BF)
                dcopy(0, j).start()

            def p1h(i, c):
                wait_a2(i)
                r = pl.multiple_of(i * 128, 128)
                v = _mlp(xrecv[pl.ds(r, 128), :], wbin[0], wbout[0]).astype(BF)
                h = _relu_mm(v, wbin[1])
                hbuf[pl.ds(r, 128), :] = h[:, HH:]
                pown[pl.ds(r, 128), :] = jnp.dot(h[:, :HH], wbout[W3O_L], preferred_element_type=F32)

                @pl.when(i == NLB - 1)
                def _():
                    with scope("s1_ol"):
                        y_wout_col(0).wait_recv()
                        orem(0)
                return c

            NA = cfg["na"]
            def p12():
                with scope("s1_p1a"):
                    lax.fori_loop(0, NA, p1, 0)
                with scope("s1_wait_w3i"):
                    y_win(1).wait_recv()
                with scope("s1_hr"):
                    hbuf[pl.ds(0, NA * 128), :] = _relu_mm(a3[pl.ds(0, NA * 128), :], wbin[W3I_R])
                with scope("s1_p1b"):
                    lax.fori_loop(NA, N1, p1h, 0)
                with scope("s1_wait_w3"):
                    y_wout_col(1).wait_recv()
                with scope("s1_p2"):
                    orem(1)
                    orem(2)
                for b in range(N1, G0):
                    with scope(f"s1_b{b}"):
                        blk(b, None)

            def blk(b, side, msgs=()):
                r = b * 128
                s = 0 if side is None else side
                wait_a2(b)
                for j in msgs:
                    dcopy(1 - s, j).wait_recv()
                if side == 1:
                    v = _mlp(xrecv[pl.ds(r, CH), :], wbin[0], wbout[0]).astype(BF)
                    v = jnp.concatenate([v, xrecv[pl.ds(r + CH, CH), :]], axis=0)
                else:
                    v = _mlp(xrecv[pl.ds(r, 128), :], wbin[0], wbout[0]).astype(BF)
                if side == 0 and b in A3:
                    a3[pl.ds(r, 128), :] = v
                else:
                    o = _mlp(v, wbin[1], wbout[1])
                    out[own(r, 128)] = o
                    ysend[pl.ds(r, 128), :] = o.astype(BF)
                for j in msgs:
                    conv_msg(1 - s, j)
                if side == 0 and b in A3:
                    acopy(BMSG[0][b][0]).start()
                else:
                    if b in GRP[s]:
                        rel_in(s, b).start()
                    for j in BMSG[s][b]:
                        dcopy(s, j).start()

            DUP = cfg.get("dup", True)
            if not DUP:
                p12()

            def p3(side):
                if DUP:
                    p12()
                for b in range(G0, 16):
                    with scope(f"s1_b{b}"):
                        blk(b, side, cfg["conv_at"][side].get(b, ()))
                if side == 1:
                    for j in A3M:
                        acopy(j).wait_recv()

            for side in cfg["ord1"]:
                pl.when(my == side)(lambda side=side: p3(side))
            with scope("s1_l3"):
                for b in A3:
                    out[0, pl.ds(b * 128, 128), :] = _mlp(a3[pl.ds(b * 128, 128), :], wbin[1], wbout[1])

            def tail(side):
                s = 1 - side
                done = [j for v in cfg["conv_at"][side].values() for j in v]
                assert len(set(done)) == len(done) and all(j in DIR[s] for j in done)
                assert not (side == 1 and any(j in A3M for j in done))
                ev = []
                rem = 0
                for j in reversed(list(DIR[s])):
                    if j not in done and not (side == 1 and j in A3M):
                        ev.append((-rem, f"d{j}"))
                    rem += DIR[s][j][1]
                rem = cfg.get("relay_early", (32, 0))[side]
                for b in reversed(list(GRP[s])):
                    ev.append((-rem, f"r{b}"))
                    rem += GRP[s][b][1]
                ev.sort()
                for _, e in ev:
                    if e not in LAST:
                        tail_ev(s, e)
                z = Z[side]
                rcopy(rows(ysend, z), rows(xrecv, z), ss.at[S_RX], xr.at[0], xnb).wait_send()

            with scope("s1_tail"):
                for slot in range(2):
                    y_win(slot, R0 * (1 - slot), DM - R0 * (1 - slot)).wait_send()
                    y_wout(slot).wait_send()
                    x_win(slot).wait_send()
                    x_wout(slot).wait_send()
                for side in cfg.get("ordt", (1, 0)):
                    pl.when(my == side)(lambda side=side: tail(side))

        if cfg.get("fin_out", True):
            for side in range(2):
                @pl.when(mx + 2 * my == 2 * side)
                def _():
                    zx = Z[1 - side]
                    rcopy(rows(xrecv, zx), rows(yrecv, zx), ss.at[S_RX], xr.at[0], xnb).wait_send()

        @pl.when(mx == 1)
        def _():
            with scope("s1_fin"):
                for e in LAST[:-1]:
                    tail_ev(0, e)
                for side in range(2):
                    @pl.when(my == side)
                    def _():
                        n = HALF - Z[side]
                        rcopy(rows(ysend, n), rows(yrecv, n), ss.at[S_Y], yr.at[0], ynb).wait_send()
                tail_ev(0, LAST[-1])

    def fn(x_padded, Win, Wout):
        return pl.pallas_call(
            body,
            out_shape=jax.ShapeDtypeStruct((1, NB, DM), F32),
            in_specs=[pl.BlockSpec(memory_space=pl.ANY)] * 3,
            out_specs=pl.BlockSpec(memory_space=pltpu.VMEM),
            scratch_shapes=[
                pltpu.VMEM((NB, DM), F32),
                pltpu.VMEM((HALF, DM), F32),
                pltpu.VMEM((2, DM, HH), F32),
                pltpu.VMEM((2, HH, DM), F32),
                pltpu.VMEM((3, DM, 2 * HH), BF),
                pltpu.VMEM((3, 2 * HH, DM), BF),
                pltpu.VMEM((HALF, DM), BF),
                pltpu.VMEM((HALF, DM), BF),
                pltpu.VMEM((HALF, DM), BF),
                pltpu.VMEM((HALF, DM), BF),
                pltpu.VMEM((P1R, HH), BF),
                pltpu.VMEM((16, HH), F32),
            ],
            compiler_params=pltpu.CompilerParams(
                collective_id=0, vmem_limit_bytes=48 * 1024 * 1024),
        )(x_padded, Win, Wout)

    return fn


_KERNEL_CFG = {}


def pallas_dist_pipemlp_pp2tp2_xy_b4096_d256_h512_kernel(x_padded, Win, Wout):
    return make(**_KERNEL_CFG)(x_padded, Win, Wout)
```

```python
import contextlib
import jax
import jax.numpy as jnp
from jax import lax
from jax.experimental import pallas as pl
from jax.experimental.pallas import tpu as pltpu

BF = jnp.bfloat16
F32 = jnp.float32
MESH = pl.DeviceIdType.MESH

NB = 4096
DM = 256
HH = 512
HALF = 2048
CH = 64
PG = 32
NPG = HALF // PG
LN = 128


def _mlp(a, win, wout):
    h = jnp.dot(a, win, preferred_element_type=F32)
    h = jnp.maximum(h, 0.0).astype(BF)
    return jnp.dot(h, wout, preferred_element_type=F32)


def _relu_mm(a, w):
    return jnp.maximum(jnp.dot(a, w, preferred_element_type=F32), 0.0).astype(BF)


def _split(total, sizes, base=0):
    out, s, i = [], 0, 0
    while s < total:
        z = min(sizes[min(i, len(sizes) - 1)], total - s)
        out.append((base + s, z))
        s += z
        i += 1
    return out


DEFAULT = dict(
    na=2,
    nl=4,
    ua=2,
    lead=4,
    rel=(((8, 128), (9, 128), (10, 96), (11, 64)),
         ((8, 128), (9, 128), (10, 96), (12, 32), (11, 64))),
    relp=(32, 48),
    a3=(12, 13),
    ev0=("i8", "i9", "x0", "i10", "x1", "x2", "i11"),
    ev1={27: ("i8",), 29: ("i9",), 31: ("i10", "x0", "i12", "i11")},
    last_split=(64, 32, 32),
    conv_at=({9: (0, 1), 12: (2,), 13: (3,), 14: (4,), 15: (7, 8, 9)},
             {10: (0, 1), 12: (2,), 13: (3,), 15: (4,)}),
    ord1=(1, 0),
    ord0=(0, 1),
    scopes=False,
)


def make(**kw):
    cfg = dict(DEFAULT)
    cfg.update(kw)
    N1 = 6
    G0 = 8
    P1R = N1 * 128
    NLB = cfg["nl"]
    NLR = NLB * 128
    UA = cfg["ua"]
    A3 = cfg["a3"]
    LEAD = cfg["lead"]
    G3 = cfg.get('g3', CH)
    NE1 = cfg.get('ne1', 7)
    NS1 = cfg.get('ns1', 5)
    LL = (8 - NE1) * 256 // G0
    RELP = ([], [])
    GRP = ({}, {})
    DIR = ({}, {})
    BMSG = ({}, {})
    Z = [0, 0]
    for s in range(2):
        for (b, n) in cfg["rel"][s]:
            idx = []
            for (a, m) in _split(n, (cfg["relp"][s],)):
                idx.append(len(RELP[s]))
                RELP[s].append((Z[s] + a, m, b * 128 + a, b))
            GRP[s][b] = (Z[s], n, b * 128, idx)
            Z[s] += n
        DIR[s][0] = (0, NLR, 0, LN)
        DIR[s][1] = (0, NLR, LN, LN)
        DIR[s][2] = (NLR, P1R - NLR, 0, DM)
        for b in range(N1, 16):
            skip = GRP[s][b][1] if b in GRP[s] else 0
            if skip == 128:
                parts = []
            elif b == 15:
                parts = _split(128 - skip, cfg["last_split"], b * 128 + skip)
            else:
                parts = [(b * 128 + skip, 128 - skip)]
            BMSG[s][b] = [3 + b - N1 + t for t in range(len(parts))]
            for key, (r, n) in zip(BMSG[s][b], parts):
                DIR[s][key] = (r, n, 0, DM)
    NREL = max(len(RELP[0]), len(RELP[1]))
    A3M = {}
    for b in A3:
        assert b not in GRP[0] and G0 <= b < 15
        A3M[BMSG[0][b][0]] = b

    KL = BMSG[0][15][-1]
    BL = cfg["rel"][0][-1][0]
    assert cfg["rel"][0][-1] == cfg["rel"][1][-1] and BMSG[0][15] == BMSG[1][15]
    LAST = [f"d{KL - 1}", f"r{BL}", f"d{KL}"]

    WINP = _split(DM, cfg.get("win_pieces", (16, 48, 32, 64, 96)))
    NPA = cfg.get("npa", 3)

    def scope(name):
        if cfg["scopes"]:
            return jax.named_scope(name)
        return contextlib.nullcontext()

    def body(x_hbm, win_hbm, wout_hbm, out,
             big, pown, wfin, wfout, wbin, wbout,
             ysend, yrecv, xsend, xrecv, hbuf, wfr):
        def scoped(ld, wr, yr, xr, ss):
            inner(x_hbm, win_hbm, wout_hbm, out, big, pown, wfin, wfout, wbin, wbout,
                  ysend, yrecv, xsend, xrecv, hbuf, wfr, ld, wr, yr, xr, ss)
        pl.run_scoped(
            scoped,
            pltpu.SemaphoreType.DMA((32,)),
            pltpu.SemaphoreType.DMA((16,)),
            pltpu.SemaphoreType.DMA((NPG + NREL,)),
            pltpu.SemaphoreType.DMA((24,)),
            pltpu.SemaphoreType.DMA((16,)),
        )

    def inner(x_hbm, win_hbm, wout_hbm, out,
              big, pown, wfin, wfout, wbin, wbout,
              ysend, yrecv, xsend, xrecv, hbuf, wfr,
              ld, wr, yr, xr, ss):
        mx = lax.axis_index("x")
        my = lax.axis_index("y")
        ynb = (mx, 1 - my)
        xnb = (1 - mx, my)
        own0 = my * HALF
        oth0 = (1 - my) * HALF
        first = mx + my == 0
        bar = pltpu.get_barrier_semaphore()

        def rcopy(src, dst, ssem, rsem, dev):
            return pltpu.make_async_remote_copy(
                src_ref=src, dst_ref=dst, send_sem=ssem, recv_sem=rsem,
                device_id=dev, device_id_type=MESH)

        hb = [1 - mx, mx]
        NP = len(WINP)
        NPRO = NP - 1
        L_WO0, L_WI1, L_WO1, L_X = NP, NP + 1, NP + 2, NP + 3

        def ld_win(slot, r0, n, k):
            return pltpu.make_async_copy(
                win_hbm.at[hb[slot], pl.ds(r0, n), :], wfin.at[slot, pl.ds(r0, n), :], ld.at[k])

        def ld_wout(slot, k):
            return pltpu.make_async_copy(wout_hbm.at[hb[slot]], wfout.at[slot], ld.at[k])

        def cv_win(slot, r0, n):
            wbin[slot, pl.ds(r0, n), pl.ds(0, HH)] = wfin[slot, pl.ds(r0, n), :].astype(BF)

        def cv_wout(slot):
            wbout[slot, pl.ds(0, HH), :] = wfout[slot].astype(BF)

        def y_win(slot, r0=0, n=DM):
            return rcopy(wbin.at[slot, pl.ds(r0, n), pl.ds(0, HH)],
                         wbin.at[slot, pl.ds(r0, n), pl.ds(HH, HH)],
                         ss.at[2 * slot], wr.at[2 * slot], ynb)

        FC = cfg.get("fc", (256, 128))
        R0 = WINP[0][1]

        def y_p0(st, part):
            c, n = ((0, FC[st]), (FC[st], HH - FC[st]))[part]
            return rcopy(wbin.at[0, pl.ds(0, R0), pl.ds(c, n)], wbin.at[0, pl.ds(0, R0), pl.ds(HH + c, n)],
                         ss.at[12 + part], wr.at[10 + part], ynb)

        def y_p0f(st):
            return rcopy(win_hbm.at[hb[0], pl.ds(0, R0), pl.ds(0, FC[st])], wfr.at[:, pl.ds(0, FC[st])],
                         ss.at[12], wr.at[10], ynb)

        def p0_recv(st):
            if FC[st]:
                @pl.when(my == 0)
                def _():
                    y_p0f(st).wait_recv()
                    y_p0(st, 0).wait_send()
                    wbin[0, pl.ds(0, R0), pl.ds(HH, FC[st])] = wfr[:, pl.ds(0, FC[st])].astype(BF)

                @pl.when(my == 1)
                def _():
                    y_p0(st, 0).wait_recv()
                    y_p0f(st).wait_send()
            y_p0(st, 1).wait()

        def y_wout(slot):
            return rcopy(wbout.at[slot, pl.ds(0, HH), :], wbout.at[slot, pl.ds(HH, HH), :],
                         ss.at[2 * slot + 1], wr.at[2 * slot + 1], ynb)

        def y_wout_col(c):
            return rcopy(wbout.at[1, pl.ds(0, HH), pl.ds(c * LN, LN)],
                         wbout.at[1, pl.ds(HH, HH), pl.ds(c * LN, LN)],
                         ss.at[3], wr.at[8 + c], ynb)

        def x_win(half, r0=0, n=DM):
            return rcopy(wbin.at[0, pl.ds(r0, n), pl.ds(half * HH, HH)],
                         wbin.at[2, pl.ds(r0, n), pl.ds(half * HH, HH)],
                         ss.at[4 + 2 * half], wr.at[4 + 2 * half], xnb)

        def x_wout(half):
            return rcopy(wbout.at[0, pl.ds(half * HH, HH), :], wbout.at[2, pl.ds(half * HH, HH), :],
                         ss.at[5 + 2 * half], wr.at[5 + 2 * half], xnb)

        S_Y, S_X, S_RY, S_RX = 8, 9, 10, 11
        RB = 1024

        def xload(i):
            base = oth0 if i % 2 == 0 else own0
            off = pl.multiple_of(base + (i // 2) * 256, 256)
            return pltpu.make_async_copy(
                x_hbm.at[0, pl.ds(off, 256), :], big.at[pl.ds(i * 256, 256), :],
                ld.at[L_X + (i // 2 if i else 8)])

        UB = cfg.get("ub", 4)
        UN = cfg.get("un", 2)
        UR = (8 - UB) * 256 // UN

        def xloadu(i):
            base = oth0 if i % 2 == 0 else own0
            off = pl.multiple_of(base + UB * 256 + (i // 2) * UR, 64)
            return pltpu.make_async_copy(
                x_hbm.at[0, pl.ds(off, UR), :], big.at[pl.ds(UB * 512 + i * UR, UR), :],
                ld.at[L_X + UB + i // 2])

        def hhalf(t, c=0):
            r = t * 256 if isinstance(t, int) else pl.multiple_of(t * 256, 256)
            pltpu.make_async_copy(
                big.at[pl.ds(r, 256), :], big.at[pl.ds(r, 256), :], ld.at[L_X + 8 * (1 - t)]).wait()
            hbuf[pl.ds(r, 256), :] = _relu_mm(big[pl.ds(r, 256), :].astype(BF), wbin[1, :, pl.ds(0, HH)])
            return c

        def rows(ref, n):
            return ref.at[pl.ds(0, n), :]

        def oth(r, n):
            return (0, pl.ds(pl.multiple_of(oth0 + r, 16), n), slice(None))

        def dcopy(s, j):
            r, n, c, nc = DIR[s][j]
            return rcopy(ysend.at[pl.ds(r, n), pl.ds(c, nc)], yrecv.at[pl.ds(r, n), pl.ds(c, nc)],
                         ss.at[S_Y], yr.at[j], ynb)

        def acopy(j):
            r, n, _, _ = DIR[0][j]
            return rcopy(xsend.at[pl.ds(r, n), :], xsend.at[pl.ds(r, n), :],
                         ss.at[S_Y], yr.at[j], ynb)

        def rel_in(s, b):
            a, n, o, _ = GRP[s][b]
            return rcopy(ysend.at[pl.ds(o, n), :], xrecv.at[pl.ds(a, n), :],
                         ss.at[S_RX], xr.at[b], xnb)

        def rel_y(s, j):
            a, n, _, _ = RELP[s][j]
            return rcopy(xrecv.at[pl.ds(a, n), :], xrecv.at[pl.ds(RB + a, n), :],
                         ss.at[S_RY], yr.at[NPG + j], ynb)

        def rel_x(s, j):
            a, n, o, b = RELP[s][j]
            return rcopy(xrecv.at[pl.ds(RB + a, n), :], yrecv.at[pl.ds(o, n), :],
                         ss.at[S_RX], xr.at[8 + b], xnb)

        def rel_xg(s, b):
            a, n, o, _ = GRP[s][b]
            return rcopy(xrecv.at[pl.ds(RB + a, n), :], yrecv.at[pl.ds(o, n), :],
                         ss.at[S_RX], xr.at[8 + b], xnb)

        def conv(r, n):
            out[oth(r, n)] = yrecv[pl.ds(r, n), :].astype(F32)

        def conv_msg(s, j):
            if j == 0:
                return
            conv(DIR[s][j][0], DIR[s][j][1])

        def tail_ev(s, e):
            j = int(e[1:])
            with scope("s1_e" + e):
                if e[0] == "d":
                    dcopy(s, j).wait_recv()
                    conv_msg(s, j)
                else:
                    rel_xg(s, j).wait_recv()
                    conv(GRP[s][j][2], GRP[s][j][1])

        def loads0(npre, lo=0, hi=99):
            def w(j):
                return lambda: ld_win(0, *WINP[j], j)

            def xl(i):
                return lambda: xload(i)
            if npre == NPRO:
                seq = [w(j) for j in range(1, npre)]
                seq += [lambda: ld_win(1, 0, DM, L_WI1), xl(0), xl(1), lambda: ld_wout(1, L_WO1)]
                seq += [w(NPRO), xl(2), xl(3), lambda: ld_wout(0, L_WO0)]
                seq += [xl(i) for i in range(4, 16)]
            else:
                if cfg.get("lo", 0) == 0:
                    seq = [lambda: ld_win(1, 0, DM, L_WI1), xl(0)]
                    seq += [w(j) for j in range(1, npre)]
                else:
                    seq = [w(j) for j in range(1, npre)]
                    seq += [lambda: ld_win(1, 0, DM, L_WI1), xl(0)]
                seq += [xl(1), lambda: ld_wout(1, L_WO1)]
                seq += [w(j) for j in range(npre, NPRO)]
                seq += [xl(2), xl(3), w(NPRO), xl(4), xl(5)]
                seq += [lambda: ld_wout(0, L_WO0)]
                seq += [xl(i) for i in range(6, 2 * UB)]
                seq += [lambda i=i: xloadu(i) for i in range(2 * UN)]
            for c in seq[lo:hi]:
                c().start()

        ST0, ST1, ST2, ST3 = cfg.get("stag", (2, 4, 6, 19))
        PRE = cfg.get("pre", 0)

        with scope("s0_pro"):
            ld_win(0, *WINP[0], 0).start()
            pl.semaphore_signal(bar, inc=1, device_id=ynb, device_id_type=MESH)

            @pl.when(mx == 0)
            def _():
                pl.semaphore_signal(bar, inc=1, device_id=xnb, device_id_type=MESH)

                @pl.when(my == 1)
                def _():
                    if FC[0]:
                        pl.semaphore_wait(bar, 1)
                        y_p0f(0).start()
                    loads0(NPRO)

                @pl.when(my == 0)
                def _():
                    loads0(NPA, 0, ST0)

            @pl.when(mx == 1)
            def _():
                seq = [lambda j=j: ld_win(0, *WINP[j], j) for j in range(1, NP)]
                seq += [lambda: ld_wout(0, L_WO0), lambda: ld_win(1, 0, DM, L_WI1), lambda: ld_wout(1, L_WO1)]
                k = cfg.get("dpre", 1)
                for c in seq[:k]:
                    c().start()
                if FC[1]:
                    @pl.when(my == 1)
                    def _():
                        pl.semaphore_wait(bar, 2)
                        y_p0f(1).start()
                for c in seq[k:]:
                    c().start()
        with scope("s0_pa"):
            ld_win(0, *WINP[0], 0).wait()
            cv_win(0, *WINP[0])

            @pl.when(first)
            def _():
                loads0(NPA, ST0, ST1)
                with scope("s0_pw"):
                    ld_win(1, 0, DM, L_WI1).wait()
                loads0(NPA, ST1, ST2)
                cv_win(1, 0, DM)
                if PRE:
                    with scope("s0_ph"):
                        hhalf(0)
                if PRE or cfg.get("p12pre", True):
                    for j in range(1, NPA):
                        ld_win(0, *WINP[j], j).wait()
                    cv_win(0, WINP[1][0], WINP[NPA][0] - WINP[1][0])
        with scope("s0_pb"):
            for st in range(2):
                @pl.when(mx == st)
                def _():
                    if FC[st]:
                        @pl.when(my == 0)
                        def _():
                            pl.semaphore_wait(bar, 1 + st)
                            y_p0(st, 0).start()
                    else:
                        pl.semaphore_wait(bar, 1 + st)
                    y_p0(st, 1).start()
        with scope("s0_pc"):
            @pl.when(first)
            def _():
                if not (PRE or cfg.get("p12pre", True)):
                    for j in range(1, NPA):
                        ld_win(0, *WINP[j], j).wait()
                    cv_win(0, WINP[1][0], WINP[NPA][0] - WINP[1][0])
                y_win(0, WINP[1][0], WINP[NPA][0] - WINP[1][0]).start()
                loads0(NPA, ST2, ST3)

            @pl.when(jnp.logical_not(first))
            def _():
                for j in range(1, NPRO):
                    ld_win(0, *WINP[j], j).wait()
                    cv_win(0, *WINP[j])
                    y_win(0, *WINP[j]).start()

        @pl.when(mx == 0)
        def _stage0():
            W0I = (1, slice(None), pl.ds(0, HH))
            W0O = (1, pl.ds(0, HH), slice(None))

            def xwait(i):
                r = i * 512 if isinstance(i, int) else pl.multiple_of(i * 512, 512)
                pltpu.make_async_copy(
                    big.at[pl.ds(r, 512), :], big.at[pl.ds(r, 512), :], ld.at[L_X + i]).wait()

            def psend(k, n=PG):
                r = k * PG if isinstance(k, int) else pl.multiple_of(k * PG, PG)
                return rcopy(ysend.at[pl.ds(r, n), :], yrecv.at[pl.ds(r, n), :],
                             ss.at[S_Y], yr.at[k], ynb)

            def pwait(r, n):
                rcopy(ysend.at[pl.ds(r, n), :], yrecv.at[pl.ds(r, n), :],
                      ss.at[S_Y], yr.at[r // PG], ynb).wait_recv()

            def psends(i):
                for q in range(8):
                    psend(i * 8 + q).start()

            def l0_out(p, r, q):
                ysend[pl.ds(q, 256), :] = p[:256].astype(BF)
                pown[pl.ds(q, 256), :] = p[256:]

            with scope("s0_init"):
                @pl.when(my == 1)
                def _():
                    ld_win(1, 0, DM, L_WI1).wait()
                    cv_win(1, 0, DM)
            with scope("s0_h0"):
                lax.fori_loop((1 - my) * PRE, 2, hhalf, 0)

                @pl.when(my == 1)
                def _():
                    ld_win(0, *WINP[NPRO], NPRO).wait()
                    cv_win(0, *WINP[NPRO])
                    y_win(0, *WINP[NPRO]).start()
                with scope("s0_hw"):
                    ld_wout(1, L_WO1).wait()
            with scope("s0_o0"):
                cv_wout(1)
                l0_out(jnp.dot(hbuf[pl.ds(0, 512), :], wbout[W0O], preferred_element_type=F32), 0, 0)

                @pl.when(my == 0)
                def _():
                    for j in range(NPA, NPRO):
                        ld_win(0, *WINP[j], j).wait()
                    cv_win(0, WINP[NPA][0], WINP[NPRO][0] - WINP[NPA][0])
                    y_win(0, WINP[NPA][0], WINP[NPRO][0] - WINP[NPA][0]).start()

            with scope("s0_l0"):
                def it(i, c):
                    r = pl.multiple_of(i * 512, 512)
                    with scope("s0_lb"):
                        with scope("s0_lx"):
                            xwait(i)
                        p = _mlp(big[pl.ds(r, 512), :].astype(BF), wbin[W0I], wbout[W0O])
                        l0_out(p, r, pl.multiple_of(i * 256, 256))
                    return c

                def ps(i, c):
                    psends(i)
                    return c

                def seg(sg, lo):
                    @pl.when(sg + 2 * my == 1)
                    def _():
                        with scope("s0_lp"):
                            ld_win(0, *WINP[NPRO], NPRO).wait()
                            cv_win(0, *WINP[NPRO])
                            y_win(0, *WINP[NPRO]).start()
                            loads0(NPA, ST3)

                    @pl.when(sg + my == 2)
                    def _():
                        with scope("s0_lw"):
                            p0_recv(0)
                            ld_wout(0, L_WO0).wait()
                            cv_wout(0)
                            y_wout(0).start()

                    @pl.when(sg + 3 * my == 2)
                    def _():
                        for k in range(LEAD):
                            psend(2 * k, CH).start()

                    @pl.when(sg + my == 3)
                    def _():
                        with scope("s0_ls"):
                            lax.fori_loop(0, NS1, ps, 0)
                    hi = jnp.where(sg == 0, 2, jnp.where(sg == 1, 3 + (NS1 - 3) * my, UB + (NE1 - UB) * my))
                    lax.fori_loop(lo, hi, it, 0)
                    return hi
                lax.fori_loop(0, 3, seg, 1)

                def itu(i, c):
                    r = pl.multiple_of(UB * 512 + i * 2 * UR, 64)
                    q = pl.multiple_of(UB * 256 + i * UR, 64)
                    with scope("s0_lu"):
                        pltpu.make_async_copy(
                            big.at[pl.ds(r, 2 * UR), :], big.at[pl.ds(r, 2 * UR), :],
                            ld.at[L_X + UB + i]).wait()
                        p = _mlp(big[pl.ds(r, 2 * UR), :].astype(BF), wbin[W0I], wbout[W0O])
                        ysend[pl.ds(q, UR), :] = p[:UR].astype(BF)
                        pown[pl.ds(q, UR), :] = p[UR:]
                    return c
                lax.fori_loop(0, UN * (1 - my), itu, 0)

            with scope("s0_wait_w1"):
                y_win(0, R0, DM - R0).wait_recv()
                y_wout(0).wait_recv()
                x_win(0).wait_recv()

            def w2wait():
                x_wout(0).wait_recv()
                x_win(1).wait_recv()
                x_wout(1).wait_recv()

            def chunk(r, n, g3=False):
                with scope("s0_wp"):
                    pwait(r, n)
                a = (pown[pl.ds(r, n), :] + yrecv[pl.ds(r, n), :].astype(F32)).astype(BF)
                a = _mlp(a, wbin[0], wbout[0]).astype(BF)
                if g3:
                    if G3 < n:
                        xsend[pl.ds(r, n - G3), :] = a[:n - G3]
                        rcopy(xsend.at[pl.ds(r, n - G3), :], xrecv.at[pl.ds(r, n - G3), :],
                              ss.at[S_X], xr.at[r // 128], xnb).start()
                        a = a[n - G3:]
                        r = pl.multiple_of(r + n - G3, 16)
                        n = G3
                    a = _mlp(a, wbin[2], wbout[2]).astype(BF)
                xsend[pl.ds(r, n), :] = a
                rcopy(xsend.at[pl.ds(r, n), :], xrecv.at[pl.ds(r, n), :],
                      ss.at[S_X], xr.at[r // 128], xnb).start()

            def relay_ev(side, ev):
                with scope("s0_" + ev):
                    j = int(ev[1:])
                    if ev[0] == "i":
                        rel_in(side, j).wait_recv()
                        for t in GRP[side][j][3]:
                            rel_y(side, t).start()
                    else:
                        rel_y(1 - side, j).wait_recv()
                        rel_x(1 - side, j).start()
                        if 1 <= j <= 8:
                            out[0, pl.ds((j - 1) * 512, 512), :] = jnp.zeros((512, DM), F32)

            def rest_ev(side, evs):
                evs = list(evs)
                rest = [f"x{j}" for j in range(len(RELP[1 - side])) if f"x{j}" not in evs]
                assert [e for e in evs if e[0] == "i"] == [f"i{b}" for b in GRP[side]]
                assert len(RELP[1 - side]) >= 9
                return rest

            def fin0(side):
                with scope("s0_fin"):
                    y_win(0, R0, DM - R0).wait_send()
                    y_wout(0).wait_send()
                    rcopy(ysend, yrecv, ss.at[S_Y], yr.at[0], ynb).wait_send()
                    rcopy(xsend, xrecv, ss.at[S_X], xr.at[0], xnb).wait_send()
                    zy, zx = Z[side], Z[1 - side]
                    rcopy(rows(xrecv, zy), rows(xrecv, zy), ss.at[S_RY], yr.at[0], ynb).wait_send()
                    if not cfg.get("fin_out", True):
                        rcopy(rows(xrecv, zx), rows(yrecv, zx), ss.at[S_RX], xr.at[0], xnb).wait_send()

            def side0():
                NIT = HALF // (PG * UA)

                def ita(j, c):
                    for u in range(UA):
                        chunk(pl.multiple_of((j * UA + u) * PG, PG), PG)

                    @pl.when(j < NIT - 2 * LEAD // UA)
                    def _():
                        for u in range(UA // 2):
                            psend(j * UA + 2 * u + 2 * LEAD, CH).start()
                    return c
                with scope("s0_p2"):
                    lax.fori_loop(0, NIT, ita, 0)
                for ev in list(cfg["ev0"]) + rest_ev(0, cfg["ev0"]):
                    relay_ev(0, ev)
                    if ev == "x0":
                        w2wait()
                fin0(0)

            def side1():
                evs = cfg["ev1"]
                rest = rest_ev(1, [e for k in sorted(evs) for e in evs[k]])
                for i in range(NS1, NE1):
                    psends(i)
                for i in range(NE1, 8):
                    xwait(i)

                def pair_late(j, c):
                    q = pl.multiple_of(NE1 * 256 + j * LL, LL)
                    rb = pl.multiple_of((q // 256) * 512 + q % 256, LL)
                    chunk(pl.multiple_of(2 * j * CH, CH), CH)
                    chunk(pl.multiple_of((2 * j + 1) * CH, CH), CH)
                    a = jnp.concatenate(
                        [big[pl.ds(rb, LL), :], big[pl.ds(pl.multiple_of(rb + 256, LL), LL), :]],
                        axis=0).astype(BF)
                    p = _mlp(a, wbin[W0I], wbout[W0O])
                    ysend[pl.ds(q, LL), :] = p[:LL].astype(BF)
                    pown[pl.ds(q, LL), :] = p[LL:]
                    for t in range(LL // PG):
                        psend(q // PG + t).start()
                    return c

                def events(j, par):
                    for k in sorted(evs):
                        if k % 2 == par and k < 31:
                            @pl.when(j == k // 2)
                            def _():
                                for ev in evs[k]:
                                    relay_ev(1, ev)

                def pair_g3(j, c):
                    chunk(pl.multiple_of(2 * j * CH, CH), CH)

                    @pl.when(j == G0)
                    def _():
                        with scope("s0_wait_w2"):
                            w2wait()
                    events(j, 0)
                    chunk(pl.multiple_of((2 * j + 1) * CH, CH), CH, True)
                    events(j, 1)
                    return c
                with scope("s0_p2a"):
                    lax.fori_loop(0, G0, pair_late, 0)
                with scope("s0_p2b"):
                    lax.fori_loop(G0, 16, pair_g3, 0)
                for ev in list(evs[31]) + rest:
                    relay_ev(1, ev)
                fin0(1)

            for side in cfg["ord0"]:
                pl.when(my == side)((side0, side1)[side])

        @pl.when(mx == 1)
        def _stage1():
            a3 = xsend
            with scope("s1_init"):
                x_win(0, 0, WINP[NPRO][0]).start()
                ld_win(0, *WINP[NPRO], NPRO).wait()
                cv_win(0, *WINP[NPRO])
                y_win(0, *WINP[NPRO]).start()
                x_win(0, *WINP[NPRO]).start()
                ld_wout(0, L_WO0).wait()
                cv_wout(0)
                y_wout(0).start()
                x_wout(0).start()
                ld_win(1, 0, DM, L_WI1).wait()
                cv_win(1, 0, DM)
                y_win(1).start()
                ld_wout(1, L_WO1).wait()
                cv_wout(1)
                y_wout_col(0).start()
                y_wout_col(1).start()
            with scope("s1_wait_w2"):
                p0_recv(1)
                y_win(0, R0, DM - R0).wait_recv()
                x_win(1).start()
                y_wout(0).wait_recv()
                x_wout(1).start()

            def wait_a2(b):
                r = b * 128 if isinstance(b, int) else pl.multiple_of(b * 128, 128)
                with scope("s1_wa"):
                    rcopy(xsend.at[pl.ds(r, 128), :], xrecv.at[pl.ds(r, 128), :],
                          ss.at[S_X], xr.at[b], xnb).wait_recv()

            def own(r, n, c=0, nc=DM):
                return (0, pl.ds(pl.multiple_of(own0 + r, 16), n), pl.ds(c, nc))

            W3I_L = (1, slice(None), pl.ds(0, HH))
            W3I_R = (1, slice(None), pl.ds(HH, HH))
            W3O_L = (1, pl.ds(0, HH), slice(None))

            def p1(i, c):
                wait_a2(i)
                r = pl.multiple_of(i * 128, 128)
                v = _mlp(xrecv[pl.ds(r, 128), :], wbin[0], wbout[0]).astype(BF)
                a3[pl.ds(r, 128), :] = v
                pown[pl.ds(r, 128), :] = _mlp(v, wbin[W3I_L], wbout[W3O_L])
                return c

            def orem(j):
                r, n, c, nc = DIR[0][j]
                o = pown[pl.ds(r, n), pl.ds(c, nc)] + jnp.dot(
                    hbuf[pl.ds(r, n), :], wbout[1, pl.ds(HH, HH), pl.ds(c, nc)],
                    preferred_element_type=F32)
                out[own(r, n, c, nc)] = o
                ysend[pl.ds(r, n), pl.ds(c, nc)] = o.astype(BF)
                dcopy(0, j).start()

            def p1h(i, c):
                wait_a2(i)
                r = pl.multiple_of(i * 128, 128)
                v = _mlp(xrecv[pl.ds(r, 128), :], wbin[0], wbout[0]).astype(BF)
                h = _relu_mm(v, wbin[1])
                hbuf[pl.ds(r, 128), :] = h[:, HH:]
                pown[pl.ds(r, 128), :] = jnp.dot(h[:, :HH], wbout[W3O_L], preferred_element_type=F32)

                @pl.when(i == NLB - 1)
                def _():
                    with scope("s1_ol"):
                        y_wout_col(0).wait_recv()
                        orem(0)
                return c

            NA = cfg["na"]
            def p12():
                with scope("s1_p1a"):
                    lax.fori_loop(0, NA, p1, 0)
                with scope("s1_wait_w3i"):
                    y_win(1).wait_recv()
                with scope("s1_hr"):
                    hbuf[pl.ds(0, NA * 128), :] = _relu_mm(a3[pl.ds(0, NA * 128), :], wbin[W3I_R])
                with scope("s1_p1b"):
                    lax.fori_loop(NA, N1, p1h, 0)
                with scope("s1_wait_w3"):
                    y_wout_col(1).wait_recv()
                with scope("s1_p2"):
                    orem(1)
                    orem(2)
                for b in range(N1, G0):
                    with scope(f"s1_b{b}"):
                        blk(b, None)

            def blk(b, side, msgs=()):
                r = b * 128
                s = 0 if side is None else side
                wait_a2(b)
                for j in msgs:
                    dcopy(1 - s, j).wait_recv()
                if side == 1:
                    v = _mlp(xrecv[pl.ds(r, 128 - G3), :], wbin[0], wbout[0]).astype(BF)
                    v = jnp.concatenate([v, xrecv[pl.ds(r + 128 - G3, G3), :]], axis=0)
                else:
                    v = _mlp(xrecv[pl.ds(r, 128), :], wbin[0], wbout[0]).astype(BF)
                if side == 0 and b in A3:
                    a3[pl.ds(r, 128), :] = v
                else:
                    o = _mlp(v, wbin[1], wbout[1])
                    out[own(r, 128)] = o
                    ysend[pl.ds(r, 128), :] = o.astype(BF)
                for j in msgs:
                    conv_msg(1 - s, j)
                if side == 0 and b in A3:
                    acopy(BMSG[0][b][0]).start()
                else:
                    if b in GRP[s]:
                        rel_in(s, b).start()
                    for j in BMSG[s][b]:
                        dcopy(s, j).start()

            DUP = cfg.get("dup", True)
            if not DUP:
                p12()

            def p3(side):
                if DUP:
                    p12()
                for b in range(G0, 16):
                    with scope(f"s1_b{b}"):
                        blk(b, side, cfg["conv_at"][side].get(b, ()))
                if side == 1:
                    for j in A3M:
                        acopy(j).wait_recv()

            for side in cfg["ord1"]:
                pl.when(my == side)(lambda side=side: p3(side))
            with scope("s1_l3"):
                for b in A3:
                    out[0, pl.ds(b * 128, 128), :] = _mlp(a3[pl.ds(b * 128, 128), :], wbin[1], wbout[1])

            def tail(side):
                s = 1 - side
                done = [j for v in cfg["conv_at"][side].values() for j in v]
                assert len(set(done)) == len(done) and all(j in DIR[s] for j in done)
                assert not (side == 1 and any(j in A3M for j in done))
                ev = []
                rem = 0
                for j in reversed(list(DIR[s])):
                    if j not in done and not (side == 1 and j in A3M):
                        ev.append((-rem, f"d{j}"))
                    rem += DIR[s][j][1]
                rem = cfg.get("relay_early", (32, 0))[side]
                for b in reversed(list(GRP[s])):
                    ev.append((-rem, f"r{b}"))
                    rem += GRP[s][b][1]
                ev.sort()
                for _, e in ev:
                    if e not in LAST:
                        tail_ev(s, e)
                z = Z[side]
                rcopy(rows(ysend, z), rows(xrecv, z), ss.at[S_RX], xr.at[0], xnb).wait_send()

            with scope("s1_tail"):
                for slot in range(2):
                    y_win(slot, R0 * (1 - slot), DM - R0 * (1 - slot)).wait_send()
                    y_wout(slot).wait_send()
                    x_win(slot).wait_send()
                    x_wout(slot).wait_send()
                for side in cfg.get("ordt", (1, 0)):
                    pl.when(my == side)(lambda side=side: tail(side))

        if cfg.get("fin_out", True):
            for side in range(2):
                @pl.when(mx + 2 * my == 2 * side)
                def _():
                    zx = Z[1 - side]
                    rcopy(rows(xrecv, zx), rows(yrecv, zx), ss.at[S_RX], xr.at[0], xnb).wait_send()

        @pl.when(mx == 1)
        def _():
            with scope("s1_fin"):
                for e in LAST[:-1]:
                    tail_ev(0, e)
                for side in range(2):
                    @pl.when(my == side)
                    def _():
                        n = HALF - Z[side]
                        rcopy(rows(ysend, n), rows(yrecv, n), ss.at[S_Y], yr.at[0], ynb).wait_send()
                tail_ev(0, LAST[-1])

    def fn(x_padded, Win, Wout):
        return pl.pallas_call(
            body,
            out_shape=jax.ShapeDtypeStruct((1, NB, DM), F32),
            in_specs=[pl.BlockSpec(memory_space=pl.ANY)] * 3,
            out_specs=pl.BlockSpec(memory_space=pltpu.VMEM),
            scratch_shapes=[
                pltpu.VMEM((NB, DM), F32),
                pltpu.VMEM((HALF, DM), F32),
                pltpu.VMEM((2, DM, HH), F32),
                pltpu.VMEM((2, HH, DM), F32),
                pltpu.VMEM((3, DM, 2 * HH), BF),
                pltpu.VMEM((3, 2 * HH, DM), BF),
                pltpu.VMEM((HALF, DM), BF),
                pltpu.VMEM((HALF, DM), BF),
                pltpu.VMEM((HALF, DM), BF),
                pltpu.VMEM((HALF, DM), BF),
                pltpu.VMEM((P1R, HH), BF),
                pltpu.VMEM((16, HH), F32),
            ],
            compiler_params=pltpu.CompilerParams(
                collective_id=0, vmem_limit_bytes=48 * 1024 * 1024),
        )(x_padded, Win, Wout)

    return fn


_KERNEL_CFG = {}


def pallas_dist_pipemlp_pp2tp2_xy_b4096_d256_h512_kernel(x_padded, Win, Wout):
    return make(**_KERNEL_CFG)(x_padded, Win, Wout)
```
